```python
import numpy as np

kernel_name = "dist_moe_top2_ep_n1024_d512_e4_h1024"

def setup_inputs():
    x = np.random.randn(1024, 512).astype(np.float32)
    router_W = np.random.randn(512, 16).astype(np.float32) * 0.1
    scores64 = x.astype(np.float64) @ router_W.astype(np.float64)
    route_idx = np.argsort(-scores64, axis=-1)[:, :2].astype(np.int32)
    expert_W = np.random.randn(16, 512, 1024).astype(np.float32) * 0.02
    return {"x": x, "router_W": router_W, "route_idx": route_idx, "expert_W": expert_W}

def reference(x, router_W, route_idx, expert_W):
    scores = x @ router_W
    s_max = scores.max(axis=-1, keepdims=True)
    probs = np.exp(scores - s_max)
    probs = probs / probs.sum(axis=-1, keepdims=True)
    out = np.zeros((1024, 1024), dtype=np.float32)
    for i in range(1024):
        e0, e1 = int(route_idx[i, 0]), int(route_idx[i, 1])
        g0, g1 = probs[i, e0], probs[i, e1]
        gs = g0 + g1
        out[i] = (g0 / gs) * (x[i] @ expert_W[e0]) + (g1 / gs) * (x[i] @ expert_W[e1])
    return out
```

```python
import contextlib

import jax
import jax.numpy as jnp
from jax import lax
from jax.experimental import pallas as pl
from jax.experimental.pallas import tpu as pltpu

N_TOK, D_MODEL, D_OUT = 1024, 512, 1024
N_DEV, N_LOCAL, N_EXP = 4, 4, 16
TM = 160
CAP = -(-(N_TOK + 16) // TM) * TM
GAP = 16
GROWS = N_TOK + GAP * 2 * N_EXP
PLANES = D_OUT // 256

BF16, F32, I32, U32 = jnp.bfloat16, jnp.float32, jnp.int32, jnp.uint32
MESH = pl.DeviceIdType.MESH
NT_DIMS = (((1,), (1,)), ((), ()))

PROFILE = False
INTERPRET = False
SCHEDULE = """
 m0 rs g0 w0b m1 m2 m3 x0a bar p0a g1 w1 x0b p0b addr c0t g2 w2
 x1 p1 c1n f0t g3 w3 c1t f1n x2 p2 c2n f1t s0t c2t x3 p3 c3n f2n s1n s1t f2t c3t
 f3n s2n s2t f3t s3n s3t
"""


def _scope(name):
    return jax.named_scope("s_" + name) if PROFILE else contextlib.nullcontext()


def _pack(lo, hi):
    lo = lax.bitcast_convert_type(lo.astype(BF16).astype(F32), U32)
    hi = lax.bitcast_convert_type(hi.astype(BF16).astype(F32), U32)
    return (lo >> 16) | hi


def _unpack(v):
    lo = lax.bitcast_convert_type(v << 16, F32)
    hi = lax.bitcast_convert_type(v & jnp.uint32(0xFFFF0000), F32)
    return lo, hi


def _iota(shape, dim):
    return lax.broadcasted_iota(I32, shape, dim)


def _onehot(cond):
    return jnp.where(cond, 1.0, 0.0).astype(BF16)


def _bucket(e, p):
    delta = (p >> 2) - (e >> 2)
    return ((p & 3) << 2) | (jnp.where((e & 1) == 1, -delta, delta) & 3)


def _lanes(v, rows):
    return jnp.concatenate(
        [jnp.broadcast_to(v[j : j + 1, :], (rows, 128)) for j in range(8)], axis=1
    )


def _sorted_pos(keys, buckets):
    n = 8 * len(buckets)
    hot = _onehot(jnp.concatenate([keys - r for r in buckets], axis=0) == 0)
    col = _iota((128, 256), 1)
    both = jnp.dot(hot, _onehot(_iota((128, 256), 0) < col), preferred_element_type=F32)
    within, total = both[:, :128], both[:, 128:]
    lower = _onehot(_iota((n, n), 1) < _iota((n, n), 0))
    base = jnp.dot(lower, total.astype(BF16), preferred_element_type=F32)
    every = within + base
    pos = jnp.full((8, 128), -1.0, F32)
    for i, r in enumerate(buckets):
        pos = jnp.where(keys == r, every[8 * i : 8 * i + 8], pos)
    return pos.astype(I32), base, base + total


def _invert(pos):
    low = _onehot(_lanes(pos & 127, 128) == _iota((128, N_TOK), 0))
    high = _lanes(pos >> 7, 8) == _iota((8, N_TOK), 0)
    t = _iota((8, N_TOK), 1)
    val = jnp.concatenate(
        [jnp.where(high, t & 127, 0), jnp.where(high, t >> 7, 0)], axis=0
    )
    inv = lax.dot_general(
        val.astype(F32).astype(BF16), low, NT_DIMS, preferred_element_type=F32
    ).astype(I32)
    return inv[:8] + (inv[8:] << 7)


def _moe_body(
    x_hbm, rw_hbm, idx_hbm, w_hbm, out_ref,
    idx_v, rw_v, w_v, xg, gate_v, part, recv, fin,
    tok_v, rs_v, addr_v, tok_s, rs_s, addr_s,
    in_sem, w_sem, meta_sem, x_sem, part_sem, fin_sem, send_sem,
):
    me = lax.axis_index("i")
    right, left = (me + 1) & 3, (me + 3) & 3

    idx_cp = pltpu.make_async_copy(idx_hbm, idx_v, in_sem.at[0])
    rw_cp = pltpu.make_async_copy(rw_hbm, rw_v, in_sem.at[1])

    w_pieces = {"0a": (0, 0, 2), "0b": (0, 2, 4), "1": (1, 0, 4), "2": (2, 0, 4), "3": (3, 0, 4)}

    def w_cp(name):
        k, s0, s1 = w_pieces[name]
        cols = pl.ds(256 * s0, 256 * (s1 - s0))
        sem = w_sem.at[list(w_pieces).index(name)]
        return pltpu.make_async_copy(w_hbm.at[k, :, cols], w_v.at[k, :, cols], sem)

    idx_cp.start()
    rw_cp.start()
    w_cp("0a").start()
    barrier = pltpu.get_barrier_semaphore()
    for d in (1, 2, 3):
        pl.semaphore_signal(barrier, inc=1, device_id=((me + d) & 3,), device_id_type=MESH)

    with _scope("idx"):
        idx_cp.wait()
    a = idx_v[pl.ds(0, 8, stride=2), :] & (N_EXP - 1)
    b = idx_v[pl.ds(1, 8, stride=2), :] & (N_EXP - 1)
    rank_ab, rank_ba = _bucket(a, b), _bucket(b, a)
    a_owns = rank_ab < ((a & 3) << 2) + 2 + (((a >> 3) ^ a ^ 1) & 1)
    owner = jnp.where(a_owns, a, b)
    rank = jnp.where(a_owns, rank_ab, rank_ba)

    n_rows, bounds = {}, {}
    sent = {"part": 0, "fin": 0, "fwd": 0}

    def tok_cp(k):
        return pltpu.make_async_copy(tok_v.at[k], tok_s.at[k], meta_sem.at[k])

    rs_cp = pltpu.make_async_copy(rs_v, rs_s, meta_sem.at[4])
    addr_cp = pltpu.make_async_copy(addr_v, addr_s, meta_sem.at[5])

    def expert_meta(k):
        e = 4 * me + k
        keys = jnp.where(a == e, rank_ab, jnp.where(b == e, rank_ba, -1))
        n_rows[k] = jnp.sum(jnp.where(keys >= 0, 1.0, 0.0)).astype(I32)
        pos, first, last = _sorted_pos(keys, range(N_EXP))
        tok_v[k] = _invert(pos)
        tok_cp(k).start()
        lane_rank = _bucket(e, _iota((1, N_EXP), 1))
        lo = hi = jnp.zeros((1, N_EXP), F32)
        for r in range(N_EXP):
            lo = jnp.where(lane_rank == r, first[8 * r : 8 * r + 1, :N_EXP], lo)
            hi = jnp.where(lane_rank == r, last[8 * r + 7 : 8 * r + 8, :N_EXP], hi)
        bounds[k] = (lo.astype(I32), hi.astype(I32))

    def bucket_starts():
        o, r = _lanes(owner, N_EXP), _lanes(rank, 32)
        sub = _iota((N_EXP, N_TOK), 0)
        lhs = jnp.concatenate([_onehot(o == sub), _onehot(o < sub)], axis=0)
        cnt = lax.dot_general(
            lhs, _onehot(r < _iota((32, N_TOK), 0)), NT_DIMS, preferred_element_type=F32
        )
        starts = cnt[:N_EXP] + cnt[N_EXP:, 16:17]
        rs_v[...] = jnp.zeros(rs_v.shape, I32)
        rs_v[:, :32] = starts.astype(I32)
        rs_cp.start()

    def out_rows():
        keys = (owner << 4) | rank
        pos = jnp.zeros((8, 128), I32)
        for c in range(N_DEV):
            for ks in ((0, 1), (2,), (3,)):
                buckets = [16 * (4 * c + k) + r for k in ks for r in range(4 * k + 3 + (len(ks) == 1))]
                p, _, _ = _sorted_pos(keys, buckets)
                pos = jnp.where(p >= 0, p + rs_s[4 * c + ks[0], 0], pos)
        t = _invert(pos)
        addr_v[...] = (((t >> 3) << 6) | (t & 7)).reshape(N_TOK)
        addr_cp.start()

    def gather(k):
        tok_cp(k).wait()

        def group(i, carry):
            for u in range(8):
                t = tok_s[k, i >> 4, ((i & 15) << 3) + u]
                pltpu.make_async_copy(
                    x_hbm.at[t >> 3, :, pl.ds(t & 7, 1), :],
                    xg.at[k, i, :, pl.ds(u, 1), :],
                    x_sem.at[k],
                ).start()
            return carry

        lax.fori_loop(0, (n_rows[k] + 7) >> 3, group, 0)

    def expert_matmul(name):
        k, s0, s1 = w_pieces[name]
        n = n_rows[k]
        with _scope("wait_x" + name):
            if s0 == 0:
                @pl.when(n > 0)
                def _():
                    rows = xg.at[k, pl.ds(0, (n + 7) >> 3)]
                    pltpu.make_async_copy(rows, rows, x_sem.at[k]).wait()
            if name == "0a":
                rw_cp.wait()
            w_cp(name).wait()

        def tile(i, carry):
            r0 = pl.multiple_of(i * TM, TM)
            xb = jnp.concatenate(
                [xg[k, pl.ds(i * (TM // 8), TM // 8), j].reshape(TM, 128) for j in range(4)],
                axis=1,
            ).astype(BF16)
            if s0 == 0:
                scores = lax.dot_general(
                    xb, rw_v[...].astype(BF16), NT_DIMS, preferred_element_type=F32
                )
                ex = jnp.exp(scores - jnp.max(scores, axis=1, keepdims=True))
                probs = ex / jnp.sum(ex, axis=1, keepdims=True)
                row = r0 + _iota((TM, N_EXP), 0)
                mine = _iota((TM, N_EXP), 1) == 4 * me + k
                other = (row >= bounds[k][0]) & (row < bounds[k][1])
                p_mine = jnp.where(mine, probs, 0.0)
                p_other = jnp.where(other, probs, 0.0)
                num = jnp.sum(p_mine + jnp.where(mine, p_other, 0.0), axis=1, keepdims=True)
                gate = num / jnp.sum(p_mine + p_other, axis=1, keepdims=True)
                gate = jnp.broadcast_to(gate, (TM, 128))
                if s1 < PLANES:
                    gate_v[pl.ds(r0, TM), :] = gate
            else:
                gate = gate_v[pl.ds(r0, TM), :]
            y = jnp.dot(
                xb, w_v[k, :, 256 * s0 : 256 * s1].astype(BF16), preferred_element_type=F32
            )
            for s in range(s0, s1):
                c = 256 * (s - s0)
                part[k, s, pl.ds(r0, TM), :] = _pack(
                    y[:, c : c + 128] * gate, y[:, c + 128 : c + 256] * gate
                )
            return carry

        lax.fori_loop(0, lax.div(n + (TM - 1), TM), tile, 0)

    def send_partials(name):
        k, s0, s1 = w_pieces[name]
        planes = pl.ds(s0, s1 - s0)
        e = 4 * me + k
        src0 = rs_s[e, 16] - rs_s[e, 0]
        for r in range(4 * k + 2, N_EXP):
            j, sub = r >> 2, r & 3
            delta = (-sub if k & 1 else sub) & 3
            dev = (me + delta) & 3
            o = 4 * dev + j
            ro = 4 * k + ((delta if j & 1 else -delta) & 3)
            first = rs_s[o, ro]
            n = rs_s[o, ro + 1] - first
            tie = int(j == k)

            @pl.when(n > 0)
            def _():
                src = part.at[k, planes, pl.ds(src0, n)]
                dst = recv.at[planes, pl.ds(first + GAP * (2 * o + tie), n)]
                sem = part_sem.at[2 * j + tie]
                if delta == 0:
                    pltpu.make_async_copy(src, dst, sem).start()
                else:
                    pltpu.make_async_remote_copy(
                        src, dst, send_sem.at[0], sem, device_id=(dev,), device_id_type=MESH
                    ).start()

            src0 = src0 + n
            if delta != 0 and s0 == 0:
                sent["part"] = sent["part"] + n

    def segment(dev, k, tie):
        e = 4 * dev + k
        first = rs_s[e, 4 * k if tie else 0]
        n = rs_s[e, 16 if tie else 4 * k] - first
        return first, first + GAP * (2 * e + tie), n, n >> 1

    def fin_rows(r0, n):
        return fin.at[pl.ds(PLANES * r0, PLANES * n)]

    def fin_send(r0, n, dev, kind, slot):
        @pl.when(n > 0)
        def _():
            rows = fin_rows(r0, n)
            pltpu.make_async_remote_copy(
                rows, rows, send_sem.at[kind], fin_sem.at[slot],
                device_id=(dev,), device_id_type=MESH,
            ).start()

    def fin_wait(r0, n, sem):
        @pl.when(n > 0)
        def _():
            rows = fin_rows(r0, n)
            pltpu.make_async_copy(rows, rows, sem).wait()

    def combine(k, tie):
        e = 4 * me + k
        first, row0, n, h = segment(me, k, tie)
        alone = rs_s[e, 4 * k + 1] - first if tie else 0

        with _scope(f"wait_c{k}{tie}"):
            @pl.when(n > alone)
            def _():
                rows = recv.at[:, pl.ds(row0 + alone, n - alone)]
                pltpu.make_async_copy(rows, rows, part_sem.at[2 * k + tie]).wait()

        src0 = first - rs_s[e, 0]

        def group(i, carry):
            for s in range(PLANES):
                theirs = recv[s, pl.ds(row0 + GAP * i, GAP), :]
                if tie:
                    theirs = jnp.where(
                        GAP * i + _iota((GAP, 128), 0) >= alone, theirs, jnp.uint32(0)
                    )
                lo0, hi0 = _unpack(part[k, s, pl.ds(src0 + GAP * i, GAP), :])
                lo1, hi1 = _unpack(theirs)
                fin[pl.ds(PLANES * (row0 + GAP * i) + s, GAP, stride=PLANES), :] = _pack(
                    lo0 + lo1, hi0 + hi1
                )
            return carry

        lax.fori_loop(0, lax.div(n + (GAP - 1), GAP), group, 0)
        q = 6 * (2 * k + tie)
        fin_send(row0, h, right, 1, q + 0)
        fin_send(row0 + h, n - h, left, 2, q + 1)
        fin_send(row0 + h, n - h, right, 1, q + 2)
        fin_send(row0, h, left, 2, q + 3)
        sent["fin"] = sent["fin"] + n

    def forward(k, tie):
        q = 6 * (2 * k + tie)
        _, row0, n, h = segment(left, k, tie)
        fin_wait(row0, h, fin_sem.at[q + 0])
        fin_send(row0, h, right, 3, q + 4)
        sent["fwd"] = sent["fwd"] + h
        _, row0, n, h = segment(right, k, tie)
        fin_wait(row0 + h, n - h, fin_sem.at[q + 1])
        fin_send(row0 + h, n - h, left, 3, q + 5)
        sent["fwd"] = sent["fwd"] + (n - h)

    def scatter_rows(first, row0, n):
        def group(i, carry):
            for u in range(8):
                p = jnp.minimum(8 * i + u, n - 1)
                v = pltpu.bitcast(fin[pl.ds(PLANES * (row0 + p), PLANES), :], BF16)
                out_ref[pl.ds(addr_s[first + p], 8, stride=8), :] = v.astype(F32)
            return carry

        lax.fori_loop(0, (n + 7) >> 3, group, 0)

    def scatter(k, tie):
        q = 6 * (2 * k + tie)
        if (k, tie) == (0, 1):
            addr_cp.wait()
        first, row0, n, h = segment(me, k, tie)
        scatter_rows(first, row0, n)
        first, row0, n, h = segment(left, k, tie)
        fin_wait(row0 + h, n - h, fin_sem.at[q + 2])
        scatter_rows(first, row0, n)
        first, row0, n, h = segment(right, k, tie)
        fin_wait(row0, h, fin_sem.at[q + 3])
        scatter_rows(first, row0, n)
        first, row0, n, h = segment((me + 2) & 3, k, tie)
        fin_wait(row0, h, fin_sem.at[q + 4])
        fin_wait(row0 + h, n - h, fin_sem.at[q + 5])
        scatter_rows(first, row0, n)

    for step in SCHEDULE.split():
        with _scope(step):
            if step == "rs":
                bucket_starts()
            elif step == "addr":
                out_rows()
            elif step == "bar":
                rs_cp.wait()
                pl.semaphore_wait(barrier, N_DEV - 1)
            elif step[0] == "m":
                expert_meta(int(step[1]))
            elif step[0] == "g":
                gather(int(step[1]))
            elif step[0] == "w":
                w_cp(step[1:]).start()
            elif step[0] == "x":
                expert_matmul(step[1:])
            elif step[0] == "p":
                send_partials(step[1:])
            else:
                {"c": combine, "f": forward, "s": scatter}[step[0]](
                    int(step[1]), int(step[2] == "t")
                )

    with _scope("drain"):
        fin_wait(0, sent["part"], send_sem.at[0])
        fin_wait(0, sent["fin"], send_sem.at[1])
        fin_wait(0, sent["fin"], send_sem.at[2])
        fin_wait(0, sent["fwd"], send_sem.at[3])


def pallas_dist_moe_top2_ep_n1024_d512_e4_h1024_kernel(x, router_W, route_idx, expert_W):
    hbm = pl.BlockSpec(memory_space=pltpu.HBM)
    dma = pltpu.SemaphoreType.DMA
    out = pl.pallas_call(
        _moe_body,
        out_shape=jax.ShapeDtypeStruct((N_TOK * 8, 128), F32),
        in_specs=[hbm] * 4,
        out_specs=pl.BlockSpec(memory_space=pltpu.VMEM),
        scratch_shapes=[
            pltpu.VMEM((16, 128), I32),
            pltpu.VMEM((N_EXP, D_MODEL), F32),
            pltpu.VMEM((N_LOCAL, D_MODEL, D_OUT), F32),
            pltpu.VMEM((N_LOCAL, CAP // 8, 4, 8, 128), F32),
            pltpu.VMEM((CAP, 128), F32),
            pltpu.VMEM((N_LOCAL, PLANES, CAP, 128), U32),
            pltpu.VMEM((PLANES, GROWS, 128), U32),
            pltpu.VMEM((PLANES * GROWS, 128), U32),
            pltpu.VMEM((N_LOCAL, 8, 128), I32),
            pltpu.VMEM((N_EXP, 128), I32),
            pltpu.VMEM((N_TOK,), I32),
            pltpu.SMEM((N_LOCAL, 8, 128), I32),
            pltpu.SMEM((N_EXP, 128), I32),
            pltpu.SMEM((N_TOK,), I32),
            dma((2,)), dma((5,)), dma((6,)), dma((N_LOCAL,)), dma((8,)), dma((48,)), dma((4,)),
        ],
        compiler_params=pltpu.CompilerParams(
            collective_id=0, vmem_limit_bytes=64 << 20, disable_bounds_checks=True
        ),
        interpret=INTERPRET,
    )(
        x.reshape(N_TOK // 8, 8, 4, 128).transpose(0, 2, 1, 3),
        router_W.T,
        route_idx.astype(I32).T.reshape(2, 8, 128).transpose(1, 0, 2).reshape(16, 128),
        expert_W,
    )
    out = out.reshape(N_TOK // 8, 8, 8, 128).transpose(0, 2, 1, 3).reshape(N_TOK, D_OUT)
    return out.astype(BF16)
```

```python
import contextlib

import jax
import jax.numpy as jnp
from jax import lax
from jax.experimental import pallas as pl
from jax.experimental.pallas import tpu as pltpu

N_TOK, D_MODEL, D_OUT = 1024, 512, 1024
N_DEV, N_LOCAL, N_EXP = 4, 4, 16
HEAD, MAIN, EXTRA = 64, 160, 64
EARLY = (8, 7, 0, 0)
GAP = 16
SEGMENTS = ((1,), (2,), (3, 4), (5, 6), (7,))
TILTED = 3

BF16, F32, I32, U32 = jnp.bfloat16, jnp.float32, jnp.int32, jnp.uint32
MESH = pl.DeviceIdType.MESH
NT_DIMS = (((1,), (1,)), ((), ()))

PROFILE = False
GUARD = True
SEM_CHECKS = False
SKEW = (0, 13, 16, 0)
HIDDEN = 65
OWN = "110000110001010010111000000111"
SCHEDULE = """
 m0 rs g0 m123 bar x00 g1 x01 G1 c00 x10 c10 g2 x11 c11 c01 G2 x20 c20 g3 x21 c21
 F1 addr f0 F0 x30 f1 x31 c30 c31 c40 c41 F2 f2 a2 F3 f3 F4 f4 a0 a1 d1 d0 a3 a4 d2 d3 d4
"""


def _scope(name):
    return jax.named_scope("s_" + name) if PROFILE else contextlib.nullcontext()


def _owns(e, p):
    (c, k), (d, j) = divmod(e, N_LOCAL), divmod(p, N_LOCAL)
    if c == d:
        return k >= j
    if k == j:
        pairs = ((0, 1), (1, 2), (2, 3), (3, 0), (0, 2), (1, 3))
        i = [set(pair) for pair in pairs].index({c, d})
        return pairs[i][1 - int(OWN[6 * k + i])] == c
    stages = ((0, 1), (0, 2), (0, 3), (1, 2), (1, 3), (2, 3))
    if ((c, d) if k < j else (d, c)) == (3, 1) and OWN[24 + stages.index((min(k, j), max(k, j)))] == "1":
        return c == 3
    return k > j


def _owns_vec(e, p):
    pair, word = (e << 4) | p, 0
    for w in range(N_EXP * N_EXP // 32):
        bits = sum(int(_owns(*divmod(32 * w + i, N_EXP))) << i for i in range(32))
        word = jnp.where(pair >> 5 == w, bits - ((bits >> 31) << 32), word)
    return ((word >> (pair & 31)) & 1) == 1


def _local_key(e, p, owned):
    delta = ((p >> 2) - (e >> 2)) & 3
    return jnp.where(owned | (delta == 0), 16, 0) | ((p & 3) << 2) | delta


def _group(k_owner, k_source):
    return 2 * max(k_owner, k_source) + int(k_source >= k_owner)


def _segment_of(group):
    return [group in groups for groups in SEGMENTS].index(True)


def _pack(lo, hi):
    lo = lax.bitcast_convert_type(lo.astype(BF16).astype(F32), U32)
    hi = lax.bitcast_convert_type(hi.astype(BF16).astype(F32), U32)
    return (lo >> 16) | hi


def _unpack(v):
    lo = lax.bitcast_convert_type(v << 16, F32)
    hi = lax.bitcast_convert_type(v & jnp.uint32(0xFFFF0000), F32)
    return lo, hi


def _iota(shape, dim):
    return lax.broadcasted_iota(I32, shape, dim)


def _ind(cond):
    return jnp.where(cond, 1.0, 0.0)


def _row(v, j, rows):
    return jnp.broadcast_to(v[j : j + 1, :], (rows, 128))


def _column_counts(keys, bound, compare):
    rows = bound.shape[0]
    return sum(_ind(compare(_row(keys, j, rows), bound)) for j in range(8)).astype(BF16)


def _total_counts(keys, bound, compare):
    counts = _column_counts(keys, bound, compare)
    return lax.dot_general(
        jnp.ones((8, 128), BF16), counts, NT_DIMS, preferred_element_type=F32
    ).astype(I32)


def _sorted_pos(keys, used, prefix):
    blocks = sorted({r // 8 for r in used})
    blocks += blocks[:1] * (len(blocks) % 2)
    bound = jnp.concatenate([8 * i + _iota((8, 128), 0) for i in blocks], axis=0)
    counts = jnp.concatenate(
        [_column_counts(keys, bound, lax.eq), _column_counts(keys, bound, lax.lt)], axis=1
    )
    before = jnp.dot(counts, prefix, preferred_element_type=F32)
    sub = _iota((8, 128), 0)
    above = sum(_ind((_row(keys, j, 8) == keys) & (sub > j)) for j in range(7))
    pos = -1.0 - above
    for r in used:
        pos = jnp.where(keys == r, _row(before, 8 * blocks.index(r // 8) + r % 8, 8), pos)
    return (pos + above).astype(I32)


def _invert(pos, rows, width):
    shift = width.bit_length() - 1
    low, val = [], []
    for j in range(8):
        low.append(_ind(_row(pos & (width - 1), j, width) == _iota((width, 128), 0)))
        high = _row(pos >> shift, j, rows) == _iota((rows, 128), 0)
        lane = _iota((rows, 128), 1).astype(F32)
        val.append(
            jnp.concatenate([jnp.where(high, lane, 0.0), jnp.where(high, float(j), 0.0)], axis=0)
        )
    inv = lax.dot_general(
        jnp.concatenate(val, axis=1).astype(BF16),
        jnp.concatenate(low, axis=1).astype(BF16),
        NT_DIMS,
        preferred_element_type=F32,
    )
    return (inv[:rows] + 128.0 * inv[rows:]).astype(I32)


def _moe_body(
    x_hbm, rw_hbm, idx_hbm, w_hbm, out_ref,
    idx_v, rw_v, w_v, xg, xb_v, gate_v, part, recv, fin, prefix_v,
    tok_v, rs_v, addr_v, tok_s, rs_s, addr_s,
    in_sem, w_sem, meta_sem, x_sem, part_sem, fin_sem, send_sem,
):
    me = lax.axis_index("i")
    right, across, left = (me + 1) & 3, (me + 2) & 3, (me + 3) & 3

    idx_cp = pltpu.make_async_copy(idx_hbm, idx_v, in_sem.at[0])
    rw_cp = pltpu.make_async_copy(rw_hbm, rw_v, in_sem.at[1])

    def w_cp(k, h):
        cols = pl.ds(512 * h, 512)
        return pltpu.make_async_copy(w_hbm.at[k, :, cols], w_v.at[k, :, cols], w_sem.at[2 * k + h])

    idx_cp.start()
    rw_cp.start()
    for k in range(N_LOCAL):
        for h in range(2):
            w_cp(k, h).start(priority=1)
    barrier = pltpu.get_barrier_semaphore()
    for dev in (right, across, left):
        pl.semaphore_signal(barrier, inc=1, device_id=(dev,), device_id_type=MESH)

    r, c = _iota((256, 128), 0), _iota((256, 128), 1)
    prefix_v[...] = _ind((r < c) | (r >= 128)).astype(BF16)
    tok_v[...] = jnp.zeros(tok_v.shape, I32)
    rs_v[...] = jnp.zeros(rs_v.shape, I32)

    with _scope("idx"):
        idx_cp.wait()
    a = idx_v[pl.ds(0, 8, stride=2), :] & (N_EXP - 1)
    b = idx_v[pl.ds(1, 8, stride=2), :] & (N_EXP - 1)
    a_owns = _owns_vec(a, b)
    key_a, key_b = _local_key(a, b, a_owns), _local_key(b, a, ~a_owns)
    owner, source = jnp.where(a_owns, a, b), jnp.where(a_owns, b, a)
    group = (
        ((owner >> 2) << 3)
        + 2 * jnp.maximum(owner & 3, source & 3)
        + jnp.where((source & 3) >= (owner & 3), 1, 0)
    )
    slot = (jnp.minimum(owner & 3, source & 3) << 2) | (((source >> 2) - (owner >> 2)) & 3)

    bounds, row_pos = {}, {}
    sent = {"fin": 0, "fwd": 0}

    def tok_cp(k, r0, rows):
        rows = pl.ds(r0, rows)
        return pltpu.make_async_copy(tok_v.at[k, rows], tok_s.at[k, rows], meta_sem.at[k])

    rs_cp = pltpu.make_async_copy(rs_v, rs_s, meta_sem.at[4])
    addr_cp = pltpu.make_async_copy(addr_v, addr_s, meta_sem.at[5])

    def bucket_start(k, key):
        return tok_s[k, 0, 64 + key]

    def expert_meta(k):
        e = 4 * me + k
        keys = jnp.where(a == e, key_a, jnp.where(b == e, key_b, 32))
        used = sorted({
            16 * int(_owns(4 * c + k, 4 * ((c + d) & 3) + j) or d == 0) + 4 * j + d
            for c in range(N_DEV) for j in range(N_LOCAL) for d in range(N_DEV)
        })
        row_pos[k] = _sorted_pos(keys, used, prefix_v[...])
        tok_v[k, :16, :16] = _invert(row_pos[k], 16, 16)
        tok_v[k, :8, 64:112] = _total_counts(keys, _iota((48, 128), 0), lax.lt)
        tok_cp(k, 0, 16).start()
        e, p = jnp.full((N_EXP, 128), e, I32), _iota((N_EXP, 128), 0)
        key = _local_key(e, p, _owns_vec(e, p))
        bounds[k] = [_total_counts(keys, key, cmp)[:1] for cmp in (lax.lt, lax.le)]

    def bucket_starts():
        g = jnp.concatenate([_row(group, j, 32) for j in range(8)], axis=1)
        s = jnp.concatenate([_row(slot, j, 32) for j in range(8)], axis=1)
        sub = _iota((32, N_TOK), 0)
        lhs = jnp.concatenate([_ind(g == sub), _ind(g < sub)], axis=0).astype(BF16)
        cnt = lax.dot_general(
            lhs, _ind(s < sub).astype(BF16), NT_DIMS, preferred_element_type=F32
        )
        rs_v[:, :32] = (cnt[:32] + cnt[32:, 16:17]).astype(I32)
        rs_cp.start()

    def out_rows():
        used = sorted({
            128 * (o >> 2) + 16 * _group(o & 3, s & 3) + 4 * min(o & 3, s & 3)
            + (((s >> 2) - (o >> 2)) & 3)
            for o in range(N_EXP) for s in range(N_EXP) if _owns(o, s)
        })
        t = _invert(_sorted_pos((group << 4) | slot, used, prefix_v[...]), 8, 128)
        addr_v[...] = (((t >> 3) << 6) | (t & 7)).reshape(N_TOK)
        addr_cp.start()

    def gather(k):
        tok_cp(k, 0, 16).wait()
        n = bucket_start(k, 32)

        @pl.when(n > 256)
        def _():
            tok_v[k, 16:, :16] = _invert(row_pos[k] - 256, 48, 16)
            tok_cp(k, 16, 48).start()
            tok_cp(k, 16, 48).wait()

        def sixteen(i, carry):
            for u in range(16):
                t = tok_s[k, i, u]
                pltpu.make_async_copy(
                    x_hbm.at[t >> 3, :, pl.ds(t & 7, 1), :],
                    xg.at[k, 2 * i + u // 8, :, pl.ds(u % 8, 1), :],
                    x_sem.at[k],
                ).start()
            return carry

        lax.fori_loop(0, (n + 15) >> 4, sixteen, 0)

    def over_extra_rows(n, fn):
        def extra(i, carry):
            fn(pl.multiple_of(MAIN + i * EXTRA, 16), EXTRA)
            return carry

        lax.fori_loop(0, lax.div(n + (EXTRA - 1 - MAIN), EXTRA), extra, 0)

    def rows_arrived(k):
        n = bucket_start(k, 32)

        @pl.when(n > 0)
        def _():
            rows = xg.at[k, pl.ds(0, 2 * ((n + 15) >> 4))]
            pltpu.make_async_copy(rows, rows, x_sem.at[k]).wait()

    def gate_tile(k, r0, m):
        xb = jnp.concatenate(
            [xg[k, pl.ds(r0 >> 3, m // 8), j].reshape(m, 128) for j in range(4)], axis=1
        ).astype(BF16)
        scores = lax.dot_general(xb, rw_v[...].astype(BF16), NT_DIMS, preferred_element_type=F32)
        ex = jnp.exp(scores - jnp.max(scores, axis=1, keepdims=True))
        probs = ex / jnp.sum(ex, axis=1, keepdims=True)
        row = r0 + _iota((m, N_EXP), 0)
        mine = _iota((m, N_EXP), 1) == 4 * me + k
        other = (row >= bounds[k][0]) & (row < bounds[k][1])
        p_mine = jnp.where(mine, probs, 0.0)
        p_other = jnp.where(other, probs, 0.0)
        num = jnp.sum(p_mine + jnp.where(mine, p_other, 0.0), axis=1, keepdims=True)
        gate = num / jnp.sum(p_mine + p_other, axis=1, keepdims=True)
        gate = jnp.broadcast_to(gate, (m, 128))
        xb_v[pl.ds(r0, m), :] = xb
        gate_v[pl.ds(r0, m), :] = gate
        return xb, gate

    gated = set()

    def gates(k):
        rows_arrived(k)
        gate_tile(k, 0, MAIN)
        over_extra_rows(bucket_start(k, 32), lambda r0, m: gate_tile(k, r0, m))
        gated.add(k)

    def expert(k, h):
        n = bucket_start(k, 32)
        fresh = k not in gated
        gated.add(k)
        with _scope(f"wait_x{k}{h}"):
            if fresh:
                rows_arrived(k)
            w_cp(k, h).wait()

        def tile(r0, m):
            if fresh:
                xb, gate = gate_tile(k, r0, m)
            else:
                xb, gate = xb_v[pl.ds(r0, m), :], gate_v[pl.ds(r0, m), :]
            y = jnp.dot(
                xb, w_v[k, :, 512 * h : 512 * h + 512].astype(BF16), preferred_element_type=F32
            )
            for s in range(2):
                part[k, h, pl.ds(2 * r0 + s, m, stride=2), :] = _pack(
                    y[:, 256 * s : 256 * s + 128] * gate, y[:, 256 * s + 128 : 256 * s + 256] * gate
                )

        sends = []
        for j in range(N_LOCAL):
            for delta in (1, 2, 3):
                if all(_owns(4 * c + k, 4 * ((c + delta) & 3) + j) for c in range(N_DEV)):
                    continue
                g, dev = _group(j, k), (me + delta) & 3
                q = _segment_of(g)
                start, end = bucket_start(k, 4 * j + delta), bucket_start(k, 4 * j + delta + 1)
                row0 = rs_s[8 * dev + g, 4 * min(j, k) + (-delta & 3)]
                row0 += GAP * (len(SEGMENTS) * dev + q)
                size = 2 * (end - start)
                now = jnp.where(end <= HEAD, size, 0) if len(sends) < EARLY[k] else 0
                sends.append((2 * start, 2 * row0, dev, q, now, size - now))

        def send(src, dst, dev, q, size):
            def start():
                pltpu.make_async_remote_copy(
                    part.at[k, h, pl.ds(src, size)],
                    recv.at[h, pl.ds(dst, size)],
                    send_sem.at[0],
                    part_sem.at[2 * q + h],
                    device_id=(dev,),
                    device_id_type=MESH,
                ).start()

            if GUARD:
                pl.when(size > 0)(start)
            else:
                start()

        if EARLY[k]:
            tile(0, HEAD)
            for *where, now, _ in sends[: EARLY[k]]:
                send(*where, now)
            tile(HEAD, MAIN - HEAD)
        else:
            tile(0, MAIN)

        over_extra_rows(n, tile)
        for *where, _, later in sends:
            send(*where, later)

    tilt = {}

    def balance():
        early = {(c, way): 0 for c in range(N_DEV) for way in (1, 3)}
        load = {
            (c, way): rs_s[8 * c + 7, 16] - rs_s[8 * c, 0] + SKEW[c]
            for c in range(N_DEV) for way in (1, 3)
        }
        for o in range(N_EXP):
            for s in range(N_EXP):
                src, delta = s >> 2, ((o >> 2) - (s >> 2)) & 3
                if delta == 0 or not _owns(o, s):
                    continue
                g, col = 8 * (o >> 2) + _group(o & 3, s & 3), 4 * min(o & 3, s & 3) + (-delta & 3)
                rows = rs_s[g, col + 1] - rs_s[g, col]
                way = delta if delta != 2 else (1 if src & 1 else 3)
                book = load if s & 3 else early
                for hop in range(2 if delta == 2 else 1):
                    book[(src + hop * way) & 3, way] += rows
        for link in load:
            load[link] += jnp.maximum(early[link] - HIDDEN, 0)
        shift = [(load[(c + 3) & 3, 3] - load[(c + 1) & 3, 1]) >> 1 for c in range(N_DEV)]
        for off in range(N_DEV):
            tilt[off] = sum(jnp.where((me + off) & 3 == c, shift[c], 0) for c in range(N_DEV))

    def segment(off, q):
        dev = (me + off) & 3
        first = rs_s[8 * dev + SEGMENTS[q][0], 0]
        n = rs_s[8 * dev + SEGMENTS[q][-1], 16] - first
        cw = (n + (q & 1)) >> 1
        if q == TILTED:
            cw = jnp.clip(cw + tilt[off], 0, n)
        return first, first + GAP * (len(SEGMENTS) * dev + q), n, cw

    def fin_send(half, r0, n, dev, kind, sem):
        @pl.when(n > 0)
        def _():
            rows = fin.at[half, pl.ds(2 * r0, 2 * n)]
            pltpu.make_async_remote_copy(
                rows, rows, send_sem.at[kind], sem, device_id=(dev,), device_id_type=MESH
            ).start()

    def fin_wait(r0, n, sem):
        @pl.when(n > 0)
        def _():
            rows = fin.at[:, pl.ds(2 * r0, 2 * n)]
            pltpu.make_async_copy(rows, rows, sem).wait()

    def combine(q, h):
        first, row0, n, cw = segment(0, q)
        pieces, alone = [], 0
        for g in SEGMENTS[q]:
            m, late = divmod(g, 2)

            def at(col, g=g):
                return rs_s[8 * me + g, col] - first

            if late:
                for k in range(m):
                    if any(_owns(e, p) for e in range(k, N_EXP, 4) for p in range(m, N_EXP, 4)):
                        pieces.append((k, 16 + 4 * m + 1, at(4 * k), at(4 * k + 4), 0))
                alone = at(4 * m + 1) - at(4 * m)
                pieces.append((m, 16 + 4 * m, at(4 * m), at(16), alone))
            else:
                pieces.append((m, 16, at(0), at(16), 0))
                for k in range(m):
                    size = at(4 * k + 1) - at(4 * k)

                    @pl.when(size > 0)
                    def _():
                        pltpu.make_async_copy(
                            part.at[k, h, pl.ds(2 * bucket_start(k, 16 + 4 * m), 2 * size)],
                            recv.at[h, pl.ds(2 * (row0 + at(4 * k)), 2 * size)],
                            part_sem.at[2 * q + h],
                        ).start()

        with _scope(f"wait_c{q}{h}"):
            @pl.when(n > alone)
            def _():
                rows = recv.at[h, pl.ds(2 * (row0 + alone), 2 * (n - alone))]
                pltpu.make_async_copy(rows, rows, part_sem.at[2 * q + h]).wait()

        for k, key, lo, hi, skip in pieces:
            src0 = bucket_start(k, key)

            def add(i, carry):
                rows = pl.ds(2 * (row0 + lo + GAP * i), 2 * GAP)
                theirs = recv[h, rows, :]
                if not isinstance(skip, int):
                    theirs = jnp.where(
                        2 * GAP * i + _iota((2 * GAP, 128), 0) >= 2 * skip, theirs, jnp.uint32(0)
                    )
                lo0, hi0 = _unpack(part[k, h, pl.ds(2 * (src0 + GAP * i), 2 * GAP), :])
                lo1, hi1 = _unpack(theirs)
                fin[h, rows, :] = _pack(lo0 + lo1, hi0 + hi1)
                return carry

            lax.fori_loop(0, lax.div(hi - lo + (GAP - 1), GAP), add, 0)

        fin_send(h, row0, cw, right, 1, fin_sem.at[6 * q + 0])
        fin_send(h, row0 + cw, n - cw, left, 2, fin_sem.at[6 * q + 1])
        fin_send(h, row0 + cw, n - cw, right, 1, fin_sem.at[6 * q + 2])
        fin_send(h, row0, cw, left, 2, fin_sem.at[6 * q + 3])
        if h == 0:
            sent["fin"] += n

    def forward_cw(q):
        _, row0, n, cw = segment(3, q)
        fin_wait(row0, cw, fin_sem.at[6 * q + 0])
        fin_send(slice(None), row0, cw, right, 3, fin_sem.at[6 * q + 4])
        sent["fwd"] += cw

    def forward_ccw(q):
        _, row0, n, cw = segment(1, q)
        fin_wait(row0 + cw, n - cw, fin_sem.at[6 * q + 1])
        fin_send(slice(None), row0 + cw, n - cw, left, 3, fin_sem.at[6 * q + 5])
        sent["fwd"] += n - cw

    addr_pending = [addr_cp]

    def scatter_rows(first, row0, n):
        if addr_pending:
            addr_pending.pop().wait()

        def put(p, count):
            lo, hi = (
                pltpu.bitcast(fin[h, pl.ds(2 * (row0 + p), 2 * count), :], BF16).astype(F32)
                for h in range(2)
            )
            for u in range(count):
                out_ref[pl.ds(addr_s[first + p + u], 8, stride=8), :] = jnp.concatenate(
                    [lo[4 * u : 4 * u + 4], hi[4 * u : 4 * u + 4]], axis=0
                )

        def sixteen(i, carry):
            put(16 * i, 16)
            return carry

        def rest(i, carry):
            for u in range(4):
                put(jnp.minimum(4 * i + u, n - 1), 1)
            return carry

        lax.fori_loop(0, n >> 4, sixteen, 0)
        lax.fori_loop((n >> 4) << 2, (n + 3) >> 2, rest, 0)

    def scatter_near(q):
        first, row0, n, cw = segment(0, q)
        scatter_rows(first, row0, n)
        first, row0, n, cw = segment(3, q)
        fin_wait(row0 + cw, n - cw, fin_sem.at[6 * q + 2])
        scatter_rows(first, row0, n)
        first, row0, n, cw = segment(1, q)
        fin_wait(row0, cw, fin_sem.at[6 * q + 3])
        scatter_rows(first, row0, n)

    def scatter_far(q):
        first, row0, n, cw = segment(2, q)
        with _scope(f"wait_d{q}cw"):
            fin_wait(row0, cw, fin_sem.at[6 * q + 4])
        with _scope(f"wait_d{q}ccw"):
            fin_wait(row0 + cw, n - cw, fin_sem.at[6 * q + 5])
        scatter_rows(first, row0, n)

    steps = {
        "g": gather, "G": gates, "x": expert, "c": combine, "f": forward_cw, "F": forward_ccw,
        "a": scatter_near, "d": scatter_far,
    }
    for step in SCHEDULE.split():
        with _scope(step):
            if step == "rs":
                bucket_starts()
            elif step == "addr":
                out_rows()
                balance()
            elif step == "bar":
                rw_cp.wait()
                rs_cp.wait()
                pl.semaphore_wait(barrier, N_DEV - 1)
            elif step[0] == "m":
                for k in step[1:]:
                    expert_meta(int(k))
            else:
                steps[step[0]](*map(int, step[1:]))

    with _scope("drain"):
        fin_wait(0, sum(bucket_start(k, 16) for k in range(N_LOCAL)), send_sem.at[0])
        fin_wait(0, sent["fin"], send_sem.at[1])
        fin_wait(0, sent["fin"], send_sem.at[2])
        fin_wait(0, sent["fwd"], send_sem.at[3])


def pallas_dist_moe_top2_ep_n1024_d512_e4_h1024_kernel(x, router_W, route_idx, expert_W):
    cap = N_TOK + EXTRA
    rows = N_TOK + GAP * N_DEV * len(SEGMENTS)
    hbm = pl.BlockSpec(memory_space=pltpu.HBM)
    dma = pltpu.SemaphoreType.DMA
    out = pl.pallas_call(
        _moe_body,
        out_shape=jax.ShapeDtypeStruct((N_TOK * 8, 128), F32),
        in_specs=[hbm] * 4,
        out_specs=pl.BlockSpec(memory_space=pltpu.VMEM),
        scratch_shapes=[
            pltpu.VMEM((16, 128), I32),
            pltpu.VMEM((N_EXP, D_MODEL), F32),
            pltpu.VMEM((N_LOCAL, D_MODEL, D_OUT), F32),
            pltpu.VMEM((N_LOCAL, cap // 8, 4, 8, 128), F32),
            pltpu.VMEM((cap, D_MODEL), BF16),
            pltpu.VMEM((cap, 128), F32),
            pltpu.VMEM((N_LOCAL, 2, 2 * cap, 128), U32),
            pltpu.VMEM((2, 2 * rows, 128), U32),
            pltpu.VMEM((2, 2 * rows, 128), U32),
            pltpu.VMEM((256, 128), BF16),
            pltpu.VMEM((N_LOCAL, 64, 128), I32),
            pltpu.VMEM((32, 128), I32),
            pltpu.VMEM((N_TOK,), I32),
            pltpu.SMEM((N_LOCAL, 64, 128), I32),
            pltpu.SMEM((32, 128), I32),
            pltpu.SMEM((N_TOK,), I32),
            dma((2,)), dma((8,)), dma((6,)), dma((N_LOCAL,)),
            dma((2 * len(SEGMENTS),)), dma((6 * len(SEGMENTS),)), dma((4,)),
        ],
        compiler_params=pltpu.CompilerParams(
            collective_id=0,
            vmem_limit_bytes=64 << 20,
            disable_bounds_checks=not SEM_CHECKS,
            disable_semaphore_checks=not SEM_CHECKS,
        ),
    )(
        x.reshape(N_TOK // 8, 8, 4, 128).transpose(0, 2, 1, 3),
        router_W.T,
        route_idx.astype(I32).T.reshape(2, 8, 128).transpose(1, 0, 2).reshape(16, 128),
        expert_W,
    )
    out = out.reshape(N_TOK // 8, 8, 8, 128).transpose(0, 2, 1, 3).reshape(N_TOK, D_OUT)
    return out.astype(BF16)
```

```python
import jax
import jax.numpy as jnp
from jax import lax
from jax.experimental import pallas as pl
from jax.experimental.pallas import tpu as pltpu

N_TOK, D_MODEL, D_OUT = 1024, 512, 1024
N_DEV, N_LOCAL, N_EXP = 4, 4, 16
CW, CCW = 1, 3

HEADS = ((64, 64), (64, 0), (0, 0), (0, 0))
HEAD_BUCKETS = 8
MAIN, EXTRA = 160, 48

SEGMENTS = ((1,), (2,), (3, 4), (5, 6), (7,))
GAP = 16

TIE_OWNER = {
    (0, 1): (0, 0, 0, 0),
    (1, 2): (1, 1, 1, 1),
    (2, 3): (3, 2, 3, 2),
    (0, 3): (0, 0, 0, 0),
    (0, 2): (2, 0, 2, 2),
    (1, 3): (3, 3, 3, 3),
}
EARLY_OWNER = ((13, 7), (14, 7))
TILTED = 3
LINK_LAG = (0, 8, 12, 0)
FREE_ROWS = 70

BF16, F32, I32, U32 = jnp.bfloat16, jnp.float32, jnp.int32, jnp.uint32
MESH = pl.DeviceIdType.MESH
NT_DIMS = (((1,), (1,)), ((), ()))


def _owns(e, p):
    (c, k), (d, j) = divmod(e, N_LOCAL), divmod(p, N_LOCAL)
    if (e, p) in EARLY_OWNER or (p, e) in EARLY_OWNER:
        return (e, p) in EARLY_OWNER
    if k == j and c != d:
        return TIE_OWNER[min(c, d), max(c, d)][k] == c
    return k >= j


def _owns_vec(e, p):
    pair, word = (e << 4) | p, 0
    for w in range(N_EXP * N_EXP // 32):
        bits = sum(int(_owns(*divmod(32 * w + i, N_EXP))) << i for i in range(32))
        word = jnp.where(pair >> 5 == w, bits - ((bits >> 31) << 32), word)
    return (word >> (pair & 31)) & 1


def _local_key(e, p, owned):
    offset = ((p >> 2) - (e >> 2)) & 3
    return (jnp.where(offset == 0, 1, owned) << 4) | ((p & 3) << 2) | offset


def _group(owner_stage, other_stage):
    return 2 * max(owner_stage, other_stage) + int(other_stage >= owner_stage)


def _global_key(o, s):
    return 8 * (o >> 2) + _group(o & 3, s & 3), 4 * min(o & 3, s & 3) + (((s >> 2) - (o >> 2)) & 3)


def _pack(lo, hi):
    lo = lax.bitcast_convert_type(lo.astype(BF16).astype(F32), U32)
    hi = lax.bitcast_convert_type(hi.astype(BF16).astype(F32), U32)
    return (lo >> 16) | hi


def _unpack(v):
    return lax.bitcast_convert_type(v << 16, F32), lax.bitcast_convert_type((v >> 16) << 16, F32)


def _iota(shape, dim):
    return lax.broadcasted_iota(I32, shape, dim)


def _ind(cond):
    return jnp.where(cond, 1.0, 0.0)


def _row(v, j, rows):
    return jnp.broadcast_to(v[j : j + 1, :], (rows, 128))


def _column_counts(keys, bound, compare):
    rows = bound.shape[0]
    return sum(_ind(compare(_row(keys, j, rows), bound)) for j in range(8)).astype(BF16)


def _sorted_pos(keys, used, prefix):
    blocks = sorted({r // 8 for r in used})
    blocks += blocks[:1] * (len(blocks) % 2)
    bound = jnp.concatenate([8 * i + _iota((8, 128), 0) for i in blocks], axis=0)
    counts = jnp.concatenate(
        [_column_counts(keys, bound, lax.eq), _column_counts(keys, bound, lax.lt)], axis=1
    )
    before = jnp.dot(counts, prefix, preferred_element_type=F32)
    sub = _iota((8, 128), 0)
    above = sum(_ind((_row(keys, j, 8) == keys) & (sub > j)) for j in range(7))
    pos = -1.0 - above
    for r in used:
        pos = jnp.where(keys == r, _row(before, 8 * blocks.index(r // 8) + r % 8, 8), pos)
    return (pos + above).astype(I32)


def _invert(pos, rows, width):
    shift = width.bit_length() - 1
    low, val = [], []
    for j in range(8):
        low.append(_ind(_row(pos & (width - 1), j, width) == _iota((width, 128), 0)))
        high = _row(pos >> shift, j, rows) == _iota((rows, 128), 0)
        lane = _iota((rows, 128), 1).astype(F32)
        val.append(
            jnp.concatenate([jnp.where(high, lane, 0.0), jnp.where(high, float(j), 0.0)], axis=0)
        )
    inv = lax.dot_general(
        jnp.concatenate(val, axis=1).astype(BF16),
        jnp.concatenate(low, axis=1).astype(BF16),
        NT_DIMS,
        preferred_element_type=F32,
    )
    return (inv[:rows] + 128.0 * inv[rows:]).astype(I32)


def _moe_body(
    x_hbm, rw_hbm, idx_hbm, w_hbm, out_ref,
    idx_v, rw_v, w_v, xg, xb_v, gate_v, part, recv, fin, prefix_v,
    tok_v, start_v, addr_v, tok_s, start_s, addr_s,
    in_sem, w_sem, meta_sem, x_sem, part_sem, hop_sem, fin_sem, send_sem,
):
    me = lax.axis_index("i")

    def chip(offset):
        return (me + offset) & 3

    def w_cp(k, h):
        cols = pl.ds(512 * h, 512)
        return pltpu.make_async_copy(w_hbm.at[k, :, cols], w_v.at[k, :, cols], w_sem.at[2 * k + h])

    def tok_cp(k, r0, rows):
        rows = pl.ds(r0, rows)
        return pltpu.make_async_copy(tok_v.at[k, rows], tok_s.at[k, rows], meta_sem.at[k])

    idx_cp = pltpu.make_async_copy(idx_hbm, idx_v, in_sem.at[0])
    rw_cp = pltpu.make_async_copy(rw_hbm, rw_v, in_sem.at[1])
    start_cp = pltpu.make_async_copy(start_v, start_s, meta_sem.at[N_LOCAL])
    addr_cp = pltpu.make_async_copy(addr_v, addr_s, meta_sem.at[N_LOCAL + 1])

    idx_cp.start()
    rw_cp.start()
    for k in range(N_LOCAL):
        for h in range(2):
            w_cp(k, h).start(priority=1)
    barrier = pltpu.get_barrier_semaphore()
    for offset in range(1, N_DEV):
        pl.semaphore_signal(barrier, inc=1, device_id=(chip(offset),), device_id_type=MESH)

    r, c = _iota((256, 128), 0), _iota((256, 128), 1)
    prefix_v[...] = _ind((r < c) | (r >= 128)).astype(BF16)
    tok_v[...] = jnp.zeros(tok_v.shape, I32)
    start_v[...] = jnp.zeros(start_v.shape, I32)
    for k in range(N_LOCAL):
        lo, hi = HEADS[k][0] // 8, MAIN // 8
        xg[k, lo:hi] = jnp.zeros((hi - lo,) + xg.shape[2:], F32)

    idx_cp.wait()
    a = idx_v[pl.ds(0, 8, stride=2), :] & (N_EXP - 1)
    b = idx_v[pl.ds(1, 8, stride=2), :] & (N_EXP - 1)
    a_owns = _owns_vec(a, b)
    key_a, key_b = _local_key(a, b, a_owns), _local_key(b, a, 1 - a_owns)
    owner, other = jnp.where(a_owns == 1, a, b), jnp.where(a_owns == 1, b, a)
    group = (
        ((owner >> 2) << 3)
        + 2 * jnp.maximum(owner & 3, other & 3)
        + jnp.where((other & 3) >= (owner & 3), 1, 0)
    )
    slot = (jnp.minimum(owner & 3, other & 3) << 2) | (((other >> 2) - (owner >> 2)) & 3)
    pairs = [(o, s) for o in range(N_EXP) for s in range(N_EXP) if _owns(o, s)]
    row_pos, partner_rows, tilt = {}, {}, {}

    def sort_expert_rows(k):
        e = 4 * me + k
        keys = jnp.where(a == e, key_a, jnp.where(b == e, key_b, 32))
        used = sorted({
            16 * int(_owns(4 * c + k, 4 * ((c + d) & 3) + j) or d == 0) + 4 * j + d
            for c in range(N_DEV) for j in range(N_LOCAL) for d in range(N_DEV)
        })
        row_pos[k] = _sorted_pos(keys, used, prefix_v[...])
        tok_v[k, :16, :16] = _invert(row_pos[k], 16, 16)
        tok_v[k, :8, 64:112] = lax.dot_general(
            jnp.ones((8, 128), BF16),
            _column_counts(keys, _iota((48, 128), 0), lax.lt),
            NT_DIMS,
            preferred_element_type=F32,
        ).astype(I32)
        tok_cp(k, 0, 16).start()
        e, p = jnp.full((N_EXP, 128), e, I32), _iota((N_EXP, 128), 0)
        key = _local_key(e, p, _owns_vec(e, p))
        partner_rows[k] = [
            jnp.dot(
                _column_counts(keys, key, compare), prefix_v[128:], preferred_element_type=F32
            ).astype(I32)
            for compare in (lax.lt, lax.le)
        ]

    def row_start(k, key):
        return tok_s[k, 0, 64 + key]

    def count_pairs():
        g = jnp.concatenate([_row(group, j, 32) for j in range(8)], axis=1)
        s = jnp.concatenate([_row(slot, j, 32) for j in range(8)], axis=1)
        sub = _iota((32, N_TOK), 0)
        lhs = jnp.concatenate([_ind(g == sub), _ind(g < sub)], axis=0).astype(BF16)
        cnt = lax.dot_general(lhs, _ind(s < sub).astype(BF16), NT_DIMS, preferred_element_type=F32)
        start_v[:, :32] = (cnt[:32] + cnt[32:, 16:17]).astype(I32)
        start_cp.start()

    def sort_tokens():
        used = sorted(16 * g + s for g, s in (_global_key(*pair) for pair in pairs))
        t = _invert(_sorted_pos((group << 4) | slot, used, prefix_v[...]), 8, 128)
        addr_v[...] = (((t >> 3) << 6) | (t & 7)).reshape(N_TOK)
        addr_cp.start()

    def balance_links():
        links = [(c, way) for c in range(N_DEV) for way in (CW, CCW)]
        early = {link: 0 for link in links}
        load = {
            (c, way): start_s[8 * c + 7, 16] - start_s[8 * c, 0] + LINK_LAG[c] for c, way in links
        }
        for o, s in pairs:
            src, offset = s >> 2, ((o >> 2) - (s >> 2)) & 3
            g, col = _global_key(o, s)
            way = offset if offset != 2 else (CW if src & 1 else CCW)
            for hop in range(min(offset, N_DEV - offset)):
                book = load if s & 3 else early
                book[(src + hop * way) & 3, way] += start_s[g, col + 1] - start_s[g, col]
        for link in links:
            load[link] += jnp.maximum(early[link] - FREE_ROWS, 0)
        shift = [(load[(c + CCW) & 3, CCW] - load[(c + CW) & 3, CW]) >> 1 for c in range(N_DEV)]
        for offset in range(N_DEV):
            tilt[offset] = sum(jnp.where(chip(offset) == c, shift[c], 0) for c in range(N_DEV))

    def extra_tiles(k):
        return lax.div(jnp.maximum(row_start(k, 32) + (EXTRA - 1 - MAIN), 0), EXTRA)

    def fetch_end(k):
        main = jnp.minimum((row_start(k, 32) + 15) >> 4, MAIN // 16)
        return main + extra_tiles(k) * (EXTRA // 16)

    def fetch_rows(k, lo, hi, sem):
        def sixteen(i, carry):
            for u in range(16):
                t = tok_s[k, i, u]
                pltpu.make_async_copy(
                    x_hbm.at[t >> 3, :, pl.ds(t & 7, 1), :],
                    xg.at[k, 2 * i + u // 8, :, pl.ds(u % 8, 1), :],
                    sem,
                ).start()
            return carry

        lax.fori_loop(lo, hi, sixteen, 0)

    def wait_rows(k, lo, hi, sem):
        rows = xg.at[k, pl.ds(2 * lo, 2 * (hi - lo))]
        pltpu.make_async_copy(rows, rows, sem).wait()

    def fetch_head(k):
        tok_cp(k, 0, 16).wait()
        fetch_rows(k, 0, HEADS[k][0] // 16, x_sem.at[2 * k])

    def fetch_body(k):
        if not HEADS[k][0]:
            tok_cp(k, 0, 16).wait()

        @pl.when(fetch_end(k) > 16)
        def _():
            tok_v[k, 16:, :16] = _invert(row_pos[k] - 256, 48, 16)
            tok_cp(k, 16, 48).start()
            tok_cp(k, 16, 48).wait()

        fetch_rows(k, HEADS[k][0] // 16, fetch_end(k), x_sem.at[2 * k + 1])

    def gate_tile(k, r0, m):
        xb = jnp.concatenate(
            [xg[k, pl.ds(r0 >> 3, m // 8), j].reshape(m, 128) for j in range(4)], axis=1
        ).astype(BF16)
        scores = lax.dot_general(rw_v[...].astype(BF16), xb, NT_DIMS, preferred_element_type=F32)
        ex = jnp.exp(scores - jnp.max(scores, axis=0, keepdims=True))
        probs = ex / jnp.sum(ex, axis=0, keepdims=True)
        row = r0 + _iota((N_EXP, m), 1)
        mine = _iota((N_EXP, m), 0) == 4 * me + k
        lo, hi = (jnp.concatenate([v] * pl.cdiv(m, 128), axis=1)[:, :m] for v in partner_rows[k])
        p_mine = jnp.where(mine, probs, 0.0)
        p_other = jnp.where((row >= lo) & (row < hi), probs, 0.0)
        share = jnp.sum(p_mine + jnp.where(mine, p_other, 0.0), axis=0, keepdims=True)
        gate = share / jnp.sum(p_mine + p_other, axis=0, keepdims=True)
        gate = jnp.broadcast_to(gate, (128, m)).T
        xb_v[pl.ds(r0, m), :] = xb
        gate_v[pl.ds(r0, m), :] = gate
        return xb, gate

    def expert_tile(k, h, r0, m):
        if h == 0:
            xb, gate = gate_tile(k, r0, m)
        else:
            xb, gate = xb_v[pl.ds(r0, m), :], gate_v[pl.ds(r0, m), :]
        w = w_v[k, :, 512 * h : 512 * h + 512].astype(BF16)
        y = jnp.dot(xb, w, preferred_element_type=F32)
        for s in range(2):
            part[k, h, pl.ds(2 * r0 + s, m, stride=2), :] = _pack(
                y[:, 256 * s : 256 * s + 128] * gate, y[:, 256 * s + 128 : 256 * s + 256] * gate
            )

    def plan_sends(k, h, head):
        targets = [
            (j, d) for j in range(N_LOCAL) for d in range(1, N_DEV)
            if not all(_owns(4 * c + k, 4 * ((c + d) & 3) + j) for c in range(N_DEV))
        ]
        plan = []
        for i, (j, d) in enumerate(targets[:HEAD_BUCKETS] if head else targets):
            g = _group(j, k)
            q = [g in groups for groups in SEGMENTS].index(True)
            lo, hi = row_start(k, 4 * j + d), row_start(k, 4 * j + d + 1)
            dst = start_s[8 * chip(d) + g, 4 * min(j, k) + (-d & 3)]
            dst += GAP * (len(SEGMENTS) * chip(d) + q)
            size = 2 * (hi - lo)
            if HEADS[k][h] and i < HEAD_BUCKETS:
                size = jnp.where(hi <= HEADS[k][h] if head else hi > HEADS[k][h], size, 0)
            plan.append((2 * lo, 2 * dst, size, chip(d), part_sem.at[2 * q + h]))
        return plan

    def send_partials(k, h, plan):
        for src, dst, size, dev, sem in plan:
            @pl.when(size > 0)
            def _():
                pltpu.make_async_remote_copy(
                    part.at[k, h, pl.ds(src, size)], recv.at[h, pl.ds(dst, size)],
                    send_sem.at[0], sem, device_id=(dev,), device_id_type=MESH,
                ).start()

    def expert_head(k, h):
        if h == 0:
            wait_rows(k, 0, HEADS[k][0] // 16, x_sem.at[2 * k])
        w_cp(k, h).wait()
        plan = plan_sends(k, h, True)
        expert_tile(k, h, 0, HEADS[k][h])
        if (k, h) == (0, 0):
            pl.semaphore_wait(barrier, N_DEV - 1)
        send_partials(k, h, plan)

    def expert_body(k, h):
        head = HEADS[k][h]
        if not head:
            w_cp(k, h).wait()
        if h == 0:
            @pl.when(fetch_end(k) > head // 16)
            def _():
                wait_rows(k, head // 16, fetch_end(k), x_sem.at[2 * k + 1])

        plan = plan_sends(k, h, False)
        expert_tile(k, h, head, MAIN - head)

        def extra(i, carry):
            expert_tile(k, h, pl.multiple_of(MAIN + i * EXTRA, 16), EXTRA)
            return carry

        lax.fori_loop(0, extra_tiles(k), extra, 0)
        send_partials(k, h, plan)

    def segment(offset, q):
        first = start_s[8 * chip(offset) + SEGMENTS[q][0], 0]
        n = start_s[8 * chip(offset) + SEGMENTS[q][-1], 16] - first
        cw = (n + (q & 1)) >> 1
        if q == TILTED:
            cw = jnp.clip(cw + tilt[offset], 0, n)
        return first, first + GAP * (len(SEGMENTS) * chip(offset) + q), n, cw

    def send_rows(h, r0, n, way, kind, sem):
        @pl.when(n > 0)
        def _():
            rows = fin.at[h, pl.ds(2 * r0, 2 * n)]
            pltpu.make_async_remote_copy(
                rows, rows, send_sem.at[kind], sem, device_id=(chip(way),), device_id_type=MESH
            ).start()

    def wait_for(buf, h, r0, n, sem):
        @pl.when(n > 0)
        def _():
            rows = buf.at[h, pl.ds(2 * r0, 2 * n)]
            pltpu.make_async_copy(rows, rows, sem).wait()

    def combine(q, h):
        first, row0, n, cw = segment(0, q)
        pieces, alone = [], 0
        for g in SEGMENTS[q]:
            m, late = divmod(g, 2)

            def at(col, g=g):
                return start_s[8 * me + g, col] - first

            if late:
                for k in range(m):
                    if any((o & 3, s & 3) == (k, m) for o, s in pairs):
                        pieces.append((k, 16 + 4 * m + 1, at(4 * k), at(4 * k + 4), False))
                alone = at(4 * m + 1) - at(4 * m)
                pieces.append((m, 16 + 4 * m, at(4 * m), at(16), True))
            else:
                pieces.append((m, 16, at(0), at(16), False))
                for k in range(m):
                    size = at(4 * k + 1) - at(4 * k)

                    @pl.when(size > 0)
                    def _():
                        pltpu.make_async_copy(
                            part.at[k, h, pl.ds(2 * row_start(k, 16 + 4 * m), 2 * size)],
                            recv.at[h, pl.ds(2 * (row0 + at(4 * k)), 2 * size)],
                            part_sem.at[2 * q + h],
                        ).start()

        wait_for(recv, h, row0 + alone, n - alone, part_sem.at[2 * q + h])
        for k, key, lo, hi, starts_alone in pieces:
            src0 = row_start(k, key)

            def add(i, carry):
                rows = pl.ds(2 * (row0 + lo + GAP * i), 2 * GAP)
                theirs = recv[h, rows, :]
                if starts_alone:
                    paired = 2 * GAP * i + _iota((2 * GAP, 128), 0) >= 2 * alone
                    theirs = jnp.where(paired, theirs, jnp.uint32(0))
                lo0, hi0 = _unpack(part[k, h, pl.ds(2 * (src0 + GAP * i), 2 * GAP), :])
                lo1, hi1 = _unpack(theirs)
                fin[h, rows, :] = _pack(lo0 + lo1, hi0 + hi1)
                return carry

            lax.fori_loop(0, lax.div(hi - lo + (GAP - 1), GAP), add, 0)

        send_rows(h, row0, cw, CW, 1, hop_sem.at[4 * q + h])
        send_rows(h, row0 + cw, n - cw, CCW, 2, hop_sem.at[4 * q + 2 + h])
        send_rows(h, row0 + cw, n - cw, CW, 1, fin_sem.at[4 * q])
        send_rows(h, row0, cw, CCW, 2, fin_sem.at[4 * q + 1])

    def passing(q, way):
        _, row0, n, cw = segment(N_DEV - way, q)
        return (row0, cw) if way == CW else (row0 + cw, n - cw)

    def forward(q, way, halves=(0, 1)):
        r0, n = passing(q, way)
        for h in halves:
            wait_for(fin, h, r0, n, hop_sem.at[4 * q + (way & 2) + h])
            send_rows(h, r0, n, way, 3, fin_sem.at[4 * q + 2 + (way >> 1)])

    def store_rows(first, row0, n):
        def put(p, count):
            lo, hi = (
                pltpu.bitcast(fin[h, pl.ds(2 * (row0 + p), 2 * count), :], BF16).astype(F32)
                for h in range(2)
            )
            for u in range(count):
                out_ref[pl.ds(addr_s[first + p + u], 8, stride=8), :] = jnp.concatenate(
                    [lo[4 * u : 4 * u + 4], hi[4 * u : 4 * u + 4]], axis=0
                )

        def sixteen(i, carry):
            put(16 * i, 16)
            return carry

        def rest(i, carry):
            for u in range(4):
                put(jnp.minimum(4 * i + u, n - 1), 1)
            return carry

        lax.fori_loop(0, n >> 4, sixteen, 0)
        lax.fori_loop((n >> 4) << 2, (n + 3) >> 2, rest, 0)

    both = slice(None)

    def store_near(q):
        first, row0, n, cw = segment(0, q)
        store_rows(first, row0, n)
        first, row0, n, cw = segment(CCW, q)
        wait_for(fin, both, row0 + cw, n - cw, fin_sem.at[4 * q])
        store_rows(first, row0, n)
        first, row0, n, cw = segment(CW, q)
        wait_for(fin, both, row0, cw, fin_sem.at[4 * q + 1])
        store_rows(first, row0, n)

    def store_far(q):
        first, row0, n, cw = segment(2, q)
        wait_for(fin, both, row0, cw, fin_sem.at[4 * q + 2])
        wait_for(fin, both, row0 + cw, n - cw, fin_sem.at[4 * q + 3])
        store_rows(first, row0, n)

    def wait_sends():
        partials = sum(row_start(k, 16) for k in range(N_LOCAL))
        owned = start_s[8 * me + 7, 16] - start_s[8 * me, 0]
        passed = sum(passing(q, way)[1] for q in range(len(SEGMENTS)) for way in (CW, CCW))
        for kind, n in enumerate((partials, owned, owned, passed)):
            wait_for(recv, both, 0, n, send_sem.at[kind])

    sort_expert_rows(0)
    count_pairs()
    fetch_head(0)
    fetch_body(0)
    sort_expert_rows(1)
    rw_cp.wait()
    start_cp.wait()
    expert_head(0, 0)
    expert_body(0, 0)
    fetch_head(1)
    expert_head(0, 1)
    expert_body(0, 1)
    combine(0, 0)
    fetch_body(1)
    sort_expert_rows(2)

    expert_head(1, 0)
    expert_body(1, 0)
    combine(1, 0)
    fetch_body(2)
    combine(0, 1)
    expert_body(1, 1)
    combine(1, 1)
    sort_expert_rows(3)
    forward(1, CCW, (0,))
    forward(1, CW, (0,))

    expert_body(2, 0)
    combine(2, 0)
    fetch_body(3)
    expert_body(2, 1)
    forward(0, CCW)
    forward(0, CW)
    combine(2, 1)
    sort_tokens()
    balance_links()
    forward(1, CCW, (1,))
    forward(1, CW, (1,))

    expert_body(3, 0)
    expert_body(3, 1)
    combine(3, 0)
    combine(3, 1)
    combine(4, 0)
    combine(4, 1)
    forward(2, CCW)
    forward(2, CW)

    addr_cp.wait()
    store_near(0)
    store_near(1)
    store_far(0)
    store_far(1)
    forward(3, CW, (0,))
    forward(3, CCW, (0,))
    store_near(2)
    forward(3, CCW, (1,))
    forward(3, CW, (1,))
    forward(4, CW)
    forward(4, CCW)
    store_near(3)
    store_near(4)
    store_far(2)
    store_far(3)
    wait_sends()
    store_far(4)


def pallas_dist_moe_top2_ep_n1024_d512_e4_h1024_kernel(
    x: jax.Array,
    router_W: jax.Array,
    route_idx: jax.Array,
    expert_W: jax.Array,
):
    cap = N_TOK + GAP
    rows = N_TOK + GAP * N_DEV * len(SEGMENTS)
    dma = pltpu.SemaphoreType.DMA
    out = pl.pallas_call(
        _moe_body,
        out_shape=jax.ShapeDtypeStruct((N_TOK * 8, 128), F32),
        in_specs=[pl.BlockSpec(memory_space=pltpu.HBM)] * 4,
        out_specs=pl.BlockSpec(memory_space=pltpu.VMEM),
        scratch_shapes=[
            pltpu.VMEM((16, 128), I32),
            pltpu.VMEM((N_EXP, D_MODEL), F32),
            pltpu.VMEM((N_LOCAL, D_MODEL, D_OUT), F32),
            pltpu.VMEM((N_LOCAL, N_TOK // 8, 4, 8, 128), F32),
            pltpu.VMEM((N_TOK, D_MODEL), BF16),
            pltpu.VMEM((N_TOK, 128), F32),
            pltpu.VMEM((N_LOCAL, 2, 2 * cap, 128), U32),
            pltpu.VMEM((2, 2 * rows, 128), U32),
            pltpu.VMEM((2, 2 * rows, 128), U32),
            pltpu.VMEM((256, 128), BF16),
            pltpu.VMEM((N_LOCAL, 64, 128), I32),
            pltpu.VMEM((32, 128), I32),
            pltpu.VMEM((N_TOK,), I32),
            pltpu.SMEM((N_LOCAL, 64, 128), I32),
            pltpu.SMEM((32, 128), I32),
            pltpu.SMEM((N_TOK,), I32),
            dma((2,)),
            dma((2 * N_LOCAL,)),
            dma((N_LOCAL + 2,)),
            dma((2 * N_LOCAL,)),
            dma((2 * len(SEGMENTS),)),
            dma((4 * len(SEGMENTS),)),
            dma((4 * len(SEGMENTS),)),
            dma((4,)),
        ],
        compiler_params=pltpu.CompilerParams(
            collective_id=0,
            vmem_limit_bytes=64 << 20,
            disable_bounds_checks=True,
            disable_semaphore_checks=True,
        ),
    )(
        x.reshape(N_TOK // 8, 8, 4, 128).transpose(0, 2, 1, 3),
        router_W.T,
        route_idx.astype(I32).T.reshape(2, 8, 128).transpose(1, 0, 2).reshape(16, 128),
        expert_W,
    )
    out = out.reshape(N_TOK // 8, 8, 8, 128).transpose(0, 2, 1, 3).reshape(N_TOK, D_OUT)
    return out.astype(BF16)
```

```python
import jax
import jax.numpy as jnp
from jax import lax
from jax.experimental import pallas as pl
from jax.experimental.pallas import tpu as pltpu

N_TOK, D_MODEL, D_OUT = 1024, 512, 1024
N_DEV, N_LOCAL, N_EXP = 4, 4, 16
CW, CCW = 1, 3

HEADS = ((64, 64), (64, 0), (0, 0), (0, 0))
HEAD_BUCKETS = 8
MAIN, EXTRA = 160, 48
assert (N_TOK - MAIN) % EXTRA == 0

SEGMENTS = ((1,), (2,), (3, 4), (5, 6), (7,))
GAP = 16

TIE_OWNER = {
    (0, 1): (0, 0, 0, 0),
    (1, 2): (1, 1, 1, 1),
    (2, 3): (3, 2, 3, 2),
    (0, 3): (0, 0, 0, 0),
    (0, 2): (2, 0, 2, 2),
    (1, 3): (3, 3, 3, 3),
}
EARLY_OWNER = ((13, 7), (14, 7))
TILTED = 3
LINK_LAG = (0, 8, 12, 0)
FREE_ROWS = 70

BF16, F32, I32, U32 = jnp.bfloat16, jnp.float32, jnp.int32, jnp.uint32
MESH = pl.DeviceIdType.MESH
NT_DIMS = (((1,), (1,)), ((), ()))


def _owns(e, p):
    (c, k), (d, j) = divmod(e, N_LOCAL), divmod(p, N_LOCAL)
    if (e, p) in EARLY_OWNER or (p, e) in EARLY_OWNER:
        return (e, p) in EARLY_OWNER
    if k == j and c != d:
        return TIE_OWNER[min(c, d), max(c, d)][k] == c
    return k >= j


def _owns_vec(e, p):
    pair, word = (e << 4) | p, 0
    for w in range(N_EXP * N_EXP // 32):
        bits = sum(int(_owns(*divmod(32 * w + i, N_EXP))) << i for i in range(32))
        word = jnp.where(pair >> 5 == w, bits - ((bits >> 31) << 32), word)
    return (word >> (pair & 31)) & 1


def _local_key(e, p, owned):
    offset = ((p >> 2) - (e >> 2)) & 3
    return (jnp.where(offset == 0, 1, owned) << 4) | ((p & 3) << 2) | offset


def _group(owner_stage, other_stage):
    return 2 * max(owner_stage, other_stage) + int(other_stage >= owner_stage)


def _global_key(o, s):
    return 8 * (o >> 2) + _group(o & 3, s & 3), 4 * min(o & 3, s & 3) + (((s >> 2) - (o >> 2)) & 3)


def _pack(lo, hi):
    lo = lax.bitcast_convert_type(lo.astype(BF16).astype(F32), U32)
    hi = lax.bitcast_convert_type(hi.astype(BF16).astype(F32), U32)
    return (lo >> 16) | hi


def _unpack(v):
    return lax.bitcast_convert_type(v << 16, F32), lax.bitcast_convert_type((v >> 16) << 16, F32)


def _split(v):
    rounded = v.astype(BF16)
    return rounded, (v - rounded.astype(F32)).astype(BF16)


def _iota(shape, dim):
    return lax.broadcasted_iota(I32, shape, dim)


def _ind(cond):
    return jnp.where(cond, 1.0, 0.0)


def _row(v, j, rows):
    return jnp.broadcast_to(v[j : j + 1, :], (rows, 128))


def _column_counts(keys, bound, compare):
    rows = bound.shape[0]
    return sum(_ind(compare(_row(keys, j, rows), bound)) for j in range(8)).astype(BF16)


def _sorted_pos(keys, used, prefix):
    blocks = sorted({r // 8 for r in used})
    blocks += blocks[:1] * (len(blocks) % 2)
    bound = jnp.concatenate([8 * i + _iota((8, 128), 0) for i in blocks], axis=0)
    counts = jnp.concatenate(
        [_column_counts(keys, bound, lax.eq), _column_counts(keys, bound, lax.lt)], axis=1
    )
    before = jnp.dot(counts, prefix, preferred_element_type=F32)
    sub = _iota((8, 128), 0)
    above = sum(_ind((_row(keys, j, 8) == keys) & (sub > j)) for j in range(7))
    pos = -1.0 - above
    for r in used:
        pos = jnp.where(keys == r, _row(before, 8 * blocks.index(r // 8) + r % 8, 8), pos)
    return (pos + above).astype(I32)


def _invert(pos, rows, width):
    shift = width.bit_length() - 1
    low, val = [], []
    for j in range(8):
        low.append(_ind(_row(pos & (width - 1), j, width) == _iota((width, 128), 0)))
        high = _row(pos >> shift, j, rows) == _iota((rows, 128), 0)
        lane = _iota((rows, 128), 1).astype(F32)
        val.append(
            jnp.concatenate([jnp.where(high, lane, 0.0), jnp.where(high, float(j), 0.0)], axis=0)
        )
    inv = lax.dot_general(
        jnp.concatenate(val, axis=1).astype(BF16),
        jnp.concatenate(low, axis=1).astype(BF16),
        NT_DIMS,
        preferred_element_type=F32,
    )
    return (inv[:rows] + 128.0 * inv[rows:]).astype(I32)


def _moe_body(
    x_hbm, rw_hbm, idx_hbm, w_hbm, out_ref,
    idx_v, rw_v, w_v, xg, xb_v, gate_v, part, recv, fin, prefix_v,
    tok_v, start_v, addr_v, tok_s, start_s, addr_s,
    in_sem, w_sem, meta_sem, x_sem, part_sem, hop_sem, fin_sem, send_sem,
):
    me = lax.axis_index("i")

    def chip(offset):
        return (me + offset) & 3

    def w_cp(k, h):
        cols = pl.ds(512 * h, 512)
        return pltpu.make_async_copy(w_hbm.at[k, :, cols], w_v.at[k, :, cols], w_sem.at[2 * k + h])

    def tok_cp(k, r0, rows):
        rows = pl.ds(r0, rows)
        return pltpu.make_async_copy(tok_v.at[k, rows], tok_s.at[k, rows], meta_sem.at[k])

    idx_cp = pltpu.make_async_copy(idx_hbm, idx_v, in_sem.at[0])
    rw_cp = pltpu.make_async_copy(rw_hbm, rw_v, in_sem.at[1])
    start_cp = pltpu.make_async_copy(start_v, start_s, meta_sem.at[N_LOCAL])
    addr_cp = pltpu.make_async_copy(addr_v, addr_s, meta_sem.at[N_LOCAL + 1])

    idx_cp.start()
    rw_cp.start()
    for k in range(N_LOCAL):
        for h in range(2):
            w_cp(k, h).start(priority=1)
    barrier = pltpu.get_barrier_semaphore()
    for offset in range(1, N_DEV):
        pl.semaphore_signal(barrier, inc=1, device_id=(chip(offset),), device_id_type=MESH)

    r, c = _iota((256, 128), 0), _iota((256, 128), 1)
    prefix_v[...] = _ind((r < c) | (r >= 128)).astype(BF16)
    tok_v[...] = jnp.zeros(tok_v.shape, I32)
    start_v[...] = jnp.zeros(start_v.shape, I32)
    for k in range(N_LOCAL):
        lo, hi = HEADS[k][0] // 8, MAIN // 8
        xg[k, lo:hi] = jnp.zeros((hi - lo,) + xg.shape[2:], F32)

    idx_cp.wait()
    a = idx_v[pl.ds(0, 8, stride=2), :] & (N_EXP - 1)
    b = idx_v[pl.ds(1, 8, stride=2), :] & (N_EXP - 1)
    a_owns = _owns_vec(a, b)
    key_a, key_b = _local_key(a, b, a_owns), _local_key(b, a, 1 - a_owns)
    owner, other = jnp.where(a_owns == 1, a, b), jnp.where(a_owns == 1, b, a)
    group = (
        ((owner >> 2) << 3)
        + 2 * jnp.maximum(owner & 3, other & 3)
        + jnp.where((other & 3) >= (owner & 3), 1, 0)
    )
    slot = (jnp.minimum(owner & 3, other & 3) << 2) | (((other >> 2) - (owner >> 2)) & 3)
    pairs = [(o, s) for o in range(N_EXP) for s in range(N_EXP) if _owns(o, s)]
    row_pos, partner_rows, tilt = {}, {}, {}

    def sort_expert_rows(k):
        e = 4 * me + k
        keys = jnp.where(a == e, key_a, jnp.where(b == e, key_b, 32))
        used = sorted({
            16 * int(_owns(4 * c + k, 4 * ((c + d) & 3) + j) or d == 0) + 4 * j + d
            for c in range(N_DEV) for j in range(N_LOCAL) for d in range(N_DEV)
        })
        row_pos[k] = _sorted_pos(keys, used, prefix_v[...])
        tok_v[k, :16, :16] = _invert(row_pos[k], 16, 16)
        tok_v[k, :8, 64:112] = lax.dot_general(
            jnp.ones((8, 128), BF16),
            _column_counts(keys, _iota((48, 128), 0), lax.lt),
            NT_DIMS,
            preferred_element_type=F32,
        ).astype(I32)
        tok_cp(k, 0, 16).start()
        e, p = jnp.full((N_EXP, 128), e, I32), _iota((N_EXP, 128), 0)
        key = _local_key(e, p, _owns_vec(e, p))
        partner_rows[k] = [
            jnp.dot(
                _column_counts(keys, key, compare), prefix_v[128:], preferred_element_type=F32
            ).astype(I32)
            for compare in (lax.lt, lax.le)
        ]

    def row_start(k, key):
        return tok_s[k, 0, 64 + key]

    def count_pairs():
        g = jnp.concatenate([_row(group, j, 32) for j in range(8)], axis=1)
        s = jnp.concatenate([_row(slot, j, 32) for j in range(8)], axis=1)
        sub = _iota((32, N_TOK), 0)
        lhs = jnp.concatenate([_ind(g == sub), _ind(g < sub)], axis=0).astype(BF16)
        cnt = lax.dot_general(lhs, _ind(s < sub).astype(BF16), NT_DIMS, preferred_element_type=F32)
        start_v[:, :32] = (cnt[:32] + cnt[32:, 16:17]).astype(I32)
        start_cp.start()

    def sort_tokens():
        used = sorted(16 * g + s for g, s in (_global_key(*pair) for pair in pairs))
        t = _invert(_sorted_pos((group << 4) | slot, used, prefix_v[...]), 8, 128)
        addr_v[...] = (((t >> 3) << 6) | (t & 7)).reshape(N_TOK)
        addr_cp.start()

    def balance_links():
        links = [(c, way) for c in range(N_DEV) for way in (CW, CCW)]
        early = {link: 0 for link in links}
        load = {
            (c, way): start_s[8 * c + 7, 16] - start_s[8 * c, 0] + LINK_LAG[c] for c, way in links
        }
        for o, s in pairs:
            src, offset = s >> 2, ((o >> 2) - (s >> 2)) & 3
            g, col = _global_key(o, s)
            way = offset if offset != 2 else (CW if src & 1 else CCW)
            for hop in range(min(offset, N_DEV - offset)):
                book = load if s & 3 else early
                book[(src + hop * way) & 3, way] += start_s[g, col + 1] - start_s[g, col]
        for link in links:
            load[link] += jnp.maximum(early[link] - FREE_ROWS, 0)
        shift = [(load[(c + CCW) & 3, CCW] - load[(c + CW) & 3, CW]) >> 1 for c in range(N_DEV)]
        for offset in range(N_DEV):
            tilt[offset] = sum(jnp.where(chip(offset) == c, shift[c], 0) for c in range(N_DEV))

    def extra_tiles(k):
        return lax.div(jnp.maximum(row_start(k, 32) + (EXTRA - 1 - MAIN), 0), EXTRA)

    def fetch_end(k):
        main = jnp.minimum((row_start(k, 32) + 15) >> 4, MAIN // 16)
        return main + extra_tiles(k) * (EXTRA // 16)

    def fetch_rows(k, lo, hi, sem):
        def sixteen(i, carry):
            for u in range(16):
                t = tok_s[k, i, u]
                pltpu.make_async_copy(
                    x_hbm.at[t >> 3, :, pl.ds(t & 7, 1), :],
                    xg.at[k, 2 * i + u // 8, :, pl.ds(u % 8, 1), :],
                    sem,
                ).start()
            return carry

        lax.fori_loop(lo, hi, sixteen, 0)

    def wait_rows(k, lo, hi, sem):
        rows = xg.at[k, pl.ds(2 * lo, 2 * (hi - lo))]
        pltpu.make_async_copy(rows, rows, sem).wait()

    def fetch_head(k):
        tok_cp(k, 0, 16).wait()
        fetch_rows(k, 0, HEADS[k][0] // 16, x_sem.at[2 * k])

    def fetch_body(k):
        if not HEADS[k][0]:
            tok_cp(k, 0, 16).wait()

        @pl.when(fetch_end(k) > 16)
        def _():
            tok_v[k, 16:, :16] = _invert(row_pos[k] - 256, 48, 16)
            tok_cp(k, 16, 48).start()
            tok_cp(k, 16, 48).wait()

        fetch_rows(k, HEADS[k][0] // 16, fetch_end(k), x_sem.at[2 * k + 1])

    def gate_tile(k, r0, m):
        xb, x_rest = _split(jnp.concatenate(
            [xg[k, pl.ds(r0 >> 3, m // 8), j].reshape(m, 128) for j in range(4)], axis=1
        ))
        rw, rw_rest = _split(rw_v[...])
        main = lax.dot_general(
            jnp.concatenate([rw, rw_rest], axis=0), xb, NT_DIMS, preferred_element_type=F32
        )
        rest = lax.dot_general(rw, x_rest, NT_DIMS, preferred_element_type=F32)
        scores = main[:N_EXP] + (main[N_EXP:] + rest)
        ex = jnp.exp(scores - jnp.max(scores, axis=0, keepdims=True))
        probs = ex / jnp.sum(ex, axis=0, keepdims=True)
        row = r0 + _iota((N_EXP, m), 1)
        mine = _iota((N_EXP, m), 0) == 4 * me + k
        lo, hi = (jnp.concatenate([v] * pl.cdiv(m, 128), axis=1)[:, :m] for v in partner_rows[k])
        p_mine = jnp.where(mine, probs, 0.0)
        p_other = jnp.where((row >= lo) & (row < hi), probs, 0.0)
        share = jnp.sum(p_mine + jnp.where(mine, p_other, 0.0), axis=0, keepdims=True)
        gate = share / jnp.sum(p_mine + p_other, axis=0, keepdims=True)
        gate = jnp.broadcast_to(gate, (128, m)).T
        xb_v[pl.ds(r0, m), :] = xb
        gate_v[pl.ds(r0, m), :] = gate
        return xb, gate

    def expert_tile(k, h, r0, m):
        if h == 0:
            xb, gate = gate_tile(k, r0, m)
        else:
            xb, gate = xb_v[pl.ds(r0, m), :], gate_v[pl.ds(r0, m), :]
        w = w_v[k, :, 512 * h : 512 * h + 512].astype(BF16)
        y = jnp.dot(xb, w, preferred_element_type=F32)
        for s in range(2):
            part[k, h, pl.ds(2 * r0 + s, m, stride=2), :] = _pack(
                y[:, 256 * s : 256 * s + 128] * gate, y[:, 256 * s + 128 : 256 * s + 256] * gate
            )

    def plan_sends(k, h, head):
        targets = [
            (j, d) for j in range(N_LOCAL) for d in range(1, N_DEV)
            if not all(_owns(4 * c + k, 4 * ((c + d) & 3) + j) for c in range(N_DEV))
        ]
        plan = []
        for i, (j, d) in enumerate(targets[:HEAD_BUCKETS] if head else targets):
            g = _group(j, k)
            q = [g in groups for groups in SEGMENTS].index(True)
            lo, hi = row_start(k, 4 * j + d), row_start(k, 4 * j + d + 1)
            dst = start_s[8 * chip(d) + g, 4 * min(j, k) + (-d & 3)]
            dst += GAP * (len(SEGMENTS) * chip(d) + q)
            size = 2 * (hi - lo)
            if HEADS[k][h] and i < HEAD_BUCKETS:
                size = jnp.where(hi <= HEADS[k][h] if head else hi > HEADS[k][h], size, 0)
            plan.append((2 * lo, 2 * dst, size, chip(d), part_sem.at[2 * q + h]))
        return plan

    def send_partials(k, h, plan):
        for src, dst, size, dev, sem in plan:
            @pl.when(size > 0)
            def _():
                pltpu.make_async_remote_copy(
                    part.at[k, h, pl.ds(src, size)], recv.at[h, pl.ds(dst, size)],
                    send_sem.at[0], sem, device_id=(dev,), device_id_type=MESH,
                ).start()

    def expert_head(k, h):
        if h == 0:
            wait_rows(k, 0, HEADS[k][0] // 16, x_sem.at[2 * k])
        w_cp(k, h).wait()
        plan = plan_sends(k, h, True)
        expert_tile(k, h, 0, HEADS[k][h])
        if (k, h) == (0, 0):
            pl.semaphore_wait(barrier, N_DEV - 1)
        send_partials(k, h, plan)

    def expert_body(k, h):
        head = HEADS[k][h]
        if not head:
            w_cp(k, h).wait()
        if h == 0:
            @pl.when(fetch_end(k) > head // 16)
            def _():
                wait_rows(k, head // 16, fetch_end(k), x_sem.at[2 * k + 1])

        plan = plan_sends(k, h, False)
        expert_tile(k, h, head, MAIN - head)

        def extra(i, carry):
            expert_tile(k, h, pl.multiple_of(MAIN + i * EXTRA, 16), EXTRA)
            return carry

        lax.fori_loop(0, extra_tiles(k), extra, 0)
        send_partials(k, h, plan)

    def segment(offset, q):
        first = start_s[8 * chip(offset) + SEGMENTS[q][0], 0]
        n = start_s[8 * chip(offset) + SEGMENTS[q][-1], 16] - first
        cw = (n + (q & 1)) >> 1
        if q == TILTED:
            cw = jnp.clip(cw + tilt[offset], 0, n)
        return first, first + GAP * (len(SEGMENTS) * chip(offset) + q), n, cw

    def send_rows(h, r0, n, way, kind, sem):
        @pl.when(n > 0)
        def _():
            rows = fin.at[h, pl.ds(2 * r0, 2 * n)]
            pltpu.make_async_remote_copy(
                rows, rows, send_sem.at[kind], sem, device_id=(chip(way),), device_id_type=MESH
            ).start()

    def wait_for(buf, h, r0, n, sem):
        @pl.when(n > 0)
        def _():
            rows = buf.at[h, pl.ds(2 * r0, 2 * n)]
            pltpu.make_async_copy(rows, rows, sem).wait()

    def combine(q, h):
        first, row0, n, cw = segment(0, q)
        pieces, alone = [], 0
        for g in SEGMENTS[q]:
            m, late = divmod(g, 2)

            def at(col, g=g):
                return start_s[8 * me + g, col] - first

            if late:
                for k in range(m):
                    if any((o & 3, s & 3) == (k, m) for o, s in pairs):
                        pieces.append((k, 16 + 4 * m + 1, at(4 * k), at(4 * k + 4), False))
                alone = at(4 * m + 1) - at(4 * m)
                pieces.append((m, 16 + 4 * m, at(4 * m), at(16), True))
            else:
                pieces.append((m, 16, at(0), at(16), False))
                for k in range(m):
                    size = at(4 * k + 1) - at(4 * k)

                    @pl.when(size > 0)
                    def _():
                        pltpu.make_async_copy(
                            part.at[k, h, pl.ds(2 * row_start(k, 16 + 4 * m), 2 * size)],
                            recv.at[h, pl.ds(2 * (row0 + at(4 * k)), 2 * size)],
                            part_sem.at[2 * q + h],
                        ).start()

        wait_for(recv, h, row0 + alone, n - alone, part_sem.at[2 * q + h])
        for k, key, lo, hi, starts_alone in pieces:
            src0 = row_start(k, key)

            def add(i, carry):
                rows = pl.ds(2 * (row0 + lo + GAP * i), 2 * GAP)
                theirs = recv[h, rows, :]
                if starts_alone:
                    paired = 2 * GAP * i + _iota((2 * GAP, 128), 0) >= 2 * alone
                    theirs = jnp.where(paired, theirs, jnp.uint32(0))
                lo0, hi0 = _unpack(part[k, h, pl.ds(2 * (src0 + GAP * i), 2 * GAP), :])
                lo1, hi1 = _unpack(theirs)
                fin[h, rows, :] = _pack(lo0 + lo1, hi0 + hi1)
                return carry

            lax.fori_loop(0, lax.div(hi - lo + (GAP - 1), GAP), add, 0)

        send_rows(h, row0, cw, CW, 1, hop_sem.at[4 * q + h])
        send_rows(h, row0 + cw, n - cw, CCW, 2, hop_sem.at[4 * q + 2 + h])
        send_rows(h, row0 + cw, n - cw, CW, 1, fin_sem.at[4 * q])
        send_rows(h, row0, cw, CCW, 2, fin_sem.at[4 * q + 1])

    def passing(q, way):
        _, row0, n, cw = segment(N_DEV - way, q)
        return (row0, cw) if way == CW else (row0 + cw, n - cw)

    def forward(q, way, halves=(0, 1)):
        r0, n = passing(q, way)
        for h in halves:
            wait_for(fin, h, r0, n, hop_sem.at[4 * q + (way & 2) + h])
            send_rows(h, r0, n, way, 3, fin_sem.at[4 * q + 2 + (way >> 1)])

    def store_rows(first, row0, n):
        def put(p, count):
            lo, hi = (
                pltpu.bitcast(fin[h, pl.ds(2 * (row0 + p), 2 * count), :], BF16).astype(F32)
                for h in range(2)
            )
            for u in range(count):
                out_ref[pl.ds(addr_s[first + p + u], 8, stride=8), :] = jnp.concatenate(
                    [lo[4 * u : 4 * u + 4], hi[4 * u : 4 * u + 4]], axis=0
                )

        def sixteen(i, carry):
            put(16 * i, 16)
            return carry

        def rest(i, carry):
            for u in range(4):
                put(jnp.minimum(4 * i + u, n - 1), 1)
            return carry

        lax.fori_loop(0, n >> 4, sixteen, 0)
        lax.fori_loop((n >> 4) << 2, (n + 3) >> 2, rest, 0)

    both = slice(None)

    def store_near(q):
        first, row0, n, cw = segment(0, q)
        store_rows(first, row0, n)
        first, row0, n, cw = segment(CCW, q)
        wait_for(fin, both, row0 + cw, n - cw, fin_sem.at[4 * q])
        store_rows(first, row0, n)
        first, row0, n, cw = segment(CW, q)
        wait_for(fin, both, row0, cw, fin_sem.at[4 * q + 1])
        store_rows(first, row0, n)

    def store_far(q):
        first, row0, n, cw = segment(2, q)
        wait_for(fin, both, row0, cw, fin_sem.at[4 * q + 2])
        wait_for(fin, both, row0 + cw, n - cw, fin_sem.at[4 * q + 3])
        store_rows(first, row0, n)

    def wait_sends():
        partials = sum(row_start(k, 16) for k in range(N_LOCAL))
        owned = start_s[8 * me + 7, 16] - start_s[8 * me, 0]
        passed = sum(passing(q, way)[1] for q in range(len(SEGMENTS)) for way in (CW, CCW))
        for kind, n in enumerate((partials, owned, owned, passed)):
            @pl.when(n > 0)
            def _():
                rows = recv.at[:, pl.ds(0, 2 * n)]
                pltpu.make_async_remote_copy(
                    rows, rows, send_sem.at[kind], part_sem.at[0],
                    device_id=(chip(CW),), device_id_type=MESH,
                ).wait_send()

    sort_expert_rows(0)
    count_pairs()
    fetch_head(0)
    fetch_body(0)
    sort_expert_rows(1)
    rw_cp.wait()
    start_cp.wait()
    expert_head(0, 0)
    expert_body(0, 0)
    fetch_head(1)
    expert_head(0, 1)
    expert_body(0, 1)
    combine(0, 0)
    fetch_body(1)
    sort_expert_rows(2)

    expert_head(1, 0)
    expert_body(1, 0)
    combine(1, 0)
    fetch_body(2)
    combine(0, 1)
    expert_body(1, 1)
    combine(1, 1)
    sort_expert_rows(3)
    forward(1, CCW, (0,))
    forward(1, CW, (0,))

    expert_body(2, 0)
    combine(2, 0)
    fetch_body(3)
    expert_body(2, 1)
    forward(0, CCW)
    forward(0, CW)
    combine(2, 1)
    sort_tokens()
    balance_links()
    forward(1, CCW, (1,))
    forward(1, CW, (1,))

    expert_body(3, 0)
    expert_body(3, 1)
    combine(3, 0)
    combine(3, 1)
    combine(4, 0)
    combine(4, 1)
    forward(2, CCW)
    forward(2, CW)

    addr_cp.wait()
    store_near(0)
    store_near(1)
    store_far(0)
    store_far(1)
    forward(3, CW, (0,))
    forward(3, CCW, (0,))
    store_near(2)
    forward(3, CCW, (1,))
    forward(3, CW, (1,))
    forward(4, CW)
    forward(4, CCW)
    store_near(3)
    store_near(4)
    store_far(2)
    store_far(3)
    wait_sends()
    store_far(4)


def pallas_dist_moe_top2_ep_n1024_d512_e4_h1024_kernel(
    x: jax.Array,
    router_W: jax.Array,
    route_idx: jax.Array,
    expert_W: jax.Array,
):
    cap = N_TOK + GAP
    rows = N_TOK + GAP * N_DEV * len(SEGMENTS)
    dma = pltpu.SemaphoreType.DMA
    out = pl.pallas_call(
        _moe_body,
        out_shape=jax.ShapeDtypeStruct((N_TOK * 8, 128), F32),
        in_specs=[pl.BlockSpec(memory_space=pltpu.HBM)] * 4,
        out_specs=pl.BlockSpec(memory_space=pltpu.VMEM),
        scratch_shapes=[
            pltpu.VMEM((16, 128), I32),
            pltpu.VMEM((N_EXP, D_MODEL), F32),
            pltpu.VMEM((N_LOCAL, D_MODEL, D_OUT), F32),
            pltpu.VMEM((N_LOCAL, N_TOK // 8, 4, 8, 128), F32),
            pltpu.VMEM((N_TOK, D_MODEL), BF16),
            pltpu.VMEM((N_TOK, 128), F32),
            pltpu.VMEM((N_LOCAL, 2, 2 * cap, 128), U32),
            pltpu.VMEM((2, 2 * rows, 128), U32),
            pltpu.VMEM((2, 2 * rows, 128), U32),
            pltpu.VMEM((256, 128), BF16),
            pltpu.VMEM((N_LOCAL, 64, 128), I32),
            pltpu.VMEM((32, 128), I32),
            pltpu.VMEM((N_TOK,), I32),
            pltpu.SMEM((N_LOCAL, 64, 128), I32),
            pltpu.SMEM((32, 128), I32),
            pltpu.SMEM((N_TOK,), I32),
            dma((2,)),
            dma((2 * N_LOCAL,)),
            dma((N_LOCAL + 2,)),
            dma((2 * N_LOCAL,)),
            dma((2 * len(SEGMENTS),)),
            dma((4 * len(SEGMENTS),)),
            dma((4 * len(SEGMENTS),)),
            dma((4,)),
        ],
        compiler_params=pltpu.CompilerParams(
            collective_id=0,
            vmem_limit_bytes=64 << 20,
            disable_bounds_checks=True,
            disable_semaphore_checks=True,
        ),
    )(
        x.reshape(N_TOK // 8, 8, 4, 128).transpose(0, 2, 1, 3),
        router_W.T,
        route_idx.astype(I32).T.reshape(2, 8, 128).transpose(1, 0, 2).reshape(16, 128),
        expert_W,
    )
    out = out.reshape(N_TOK // 8, 8, 8, 128).transpose(0, 2, 1, 3).reshape(N_TOK, D_OUT)
    return out.astype(BF16)
```
